```python
import numpy as np

kernel_name = "dist_sparse_attn_localglobal_qseq_kvseq_b2_sq128_skv128_hq4_dh64"

def setup_inputs():
    x = np.random.randn(2, 512, 512).astype(np.float32)
    Wq = np.random.randn(512, 256).astype(np.float32) * 0.02
    K_ext = np.random.randn(2, 512, 4, 64).astype(np.float32)
    V_ext = np.random.randn(2, 512, 4, 64).astype(np.float32)
    Wo = np.random.randn(256, 512).astype(np.float32) * 0.02
    return {"x": x, "Wq": Wq, "K_ext": K_ext, "V_ext": V_ext, "Wo": Wo}

def reference(x, Wq, K_ext, V_ext, Wo):
    B, Sq, Skv, Hq, Dh = 2, 512, 512, 4, 64
    Q = (x @ Wq).reshape(B, Sq, Hq, Dh)
    qi = np.arange(Sq)[:, None]
    ki = np.arange(Skv)[None, :]
    local = np.abs(qi - ki) <= 128
    glob = (ki < 32) | (qi < 32)
    mask = local | glob
    scores = np.einsum('bihd,bjhd->bhij', Q, K_ext).astype(np.float32) * 0.125
    scores = np.where(mask[None, None, :, :], scores, -1e9)
    scores_max = scores.max(axis=-1, keepdims=True)
    w = np.exp(scores - scores_max)
    row_keep = mask.any(axis=1)
    w_sum = np.where(row_keep[None, None, :, None], w.sum(axis=-1, keepdims=True), 1.0)
    w = w / w_sum
    w = np.where(row_keep[None, None, :, None], w, 0.0)
    ctx = np.einsum('bhij,bjhd->bihd', w, V_ext).reshape(B, Sq, Hq * Dh)
    return ctx @ Wo
```

```python
import functools
import jax
import jax.numpy as jnp
from jax import lax
from jax.experimental import pallas as pl
from jax.experimental.pallas import tpu as pltpu

MESH = pl.DeviceIdType.MESH
F32 = jnp.float32
BF16 = jnp.bfloat16
NEG = -1e30
LOG2E = 1.4426950408889634
T = 128
NG = 4


def pallas_dist_sparse_attn_localglobal_qseq_kvseq_b2_sq128_skv128_hq4_dh64_kernel(x, Wq, K_ext, V_ext, Wo):
    kt = jnp.transpose(K_ext, (0, 2, 3, 1)).reshape(512, 128)
    vt = jnp.transpose(V_ext, (0, 2, 3, 1)).reshape(512, 128)
    x2 = x.reshape(256, 512)

    def body(x_hbm, wq_hbm, kt_hbm, vt_hbm, wo_hbm, out_ref,
             x32, wq32, wo32, kv32, kvb, kvL, kvR, kvg, qp, qg, gctx1, glse1, gctx3, glse3,
             lsem, ssem, rsemL, rsemR, rsemG, ready):
        my = lax.axis_index("i")
        bar = pltpu.get_barrier_semaphore()

        lane = lax.broadcasted_iota(jnp.int32, (T, T), 1)
        lo = lane < 64
        lane2 = lax.broadcasted_iota(jnp.int32, (2 * T, T), 1)
        row2 = lax.broadcasted_iota(jnp.int32, (2 * T, T), 0) & (T - 1)
        lane_g = lax.broadcasted_iota(jnp.int32, (32, T), 1)
        lo_g = lane_g < 64

        def signal(sem, to):
            pl.semaphore_signal(sem, inc=1, device_id=(to,), device_id_type=MESH)

        def kv_load(kind, g):
            src = (kt_hbm, vt_hbm)[kind]
            return pltpu.make_async_copy(src.at[pl.ds(g * T, T)], kv32.at[kind, g], lsem.at[kind * 4 + g])

        ld_x = pltpu.make_async_copy(x_hbm, x32, lsem.at[8])
        ld_wq = pltpu.make_async_copy(wq_hbm, wq32, lsem.at[9])
        ld_wo = pltpu.make_async_copy(wo_hbm, wo32, lsem.at[10])

        def rdma(src, dst, s, r, to):
            return pltpu.make_async_remote_copy(src, dst, s, r, device_id=(to,), device_id_type=MESH)

        def stack(tile, lo_mask):
            z = jnp.zeros_like(tile)
            return jnp.concatenate([jnp.where(lo_mask, tile, z), jnp.where(lo_mask, z, tile)], axis=0)

        def dot_nn(a, b):
            return jnp.dot(a, b, preferred_element_type=F32)

        def dot_nt(a, b):
            return lax.dot_general(a, b, (((1,), (1,)), ((), ())), preferred_element_type=F32)

        def softmax_parts(q2, blocks):
            ss = []
            for k_tile, mask in blocks:
                s = dot_nn(q2, k_tile)
                if mask is not None:
                    s = jnp.where(mask, s, NEG)
                ss.append(s)
            m = functools.reduce(jnp.maximum, ss)
            m = jnp.max(m, axis=1, keepdims=True)
            ps = [jnp.exp2(s - m) for s in ss]
            l = jnp.sum(functools.reduce(jnp.add, ps), axis=1, keepdims=True)
            return [p.astype(BF16) for p in ps], m, l

        def unstack(o, lo_mask):
            n = o.shape[0] // 2
            return jnp.where(lo_mask, jnp.broadcast_to(o[:n], (n, T)), jnp.broadcast_to(o[n:], (n, T)))

        def program(p):
            has_left = p > 0
            has_right = p < 3
            order = {0: (2, 3, 0, 1), 1: (0, 1, 2, 3), 2: (0, 1, 2, 3), 3: (0, 1, 2, 3)}[p]
            proc = {0: (0, 1, 2, 3), 1: (2, 3, 0, 1), 2: (0, 1, 2, 3), 3: (0, 1, 2, 3)}[p]
            if p == 0:
                signal(bar, 1); signal(bar, 3)
            elif p == 1:
                signal(bar, 0); signal(bar, 2)
            elif p == 2:
                signal(bar, 3)
            else:
                signal(bar, 0); signal(bar, 2)
            if p == 2:
                order = (0, 2, 1, 3)
            if p == 0:
                ld_wq.start(); ld_x.start()
            for g in order:
                kv_load(0, g).start(); kv_load(1, g).start()
            if p != 0:
                ld_x.start(); ld_wq.start()
            ld_wo.start()

            sends = []

            def send(src, dst, rsem, to):
                c = rdma(src, dst, ssem.at[len(sends)], rsem, to)
                c.start()
                sends.append(c)

            def recv(dst, rsem):
                rdma(dst, dst, ssem.at[0], rsem, 0).wait_recv()

            def convert(kind, g):
                kv_load(kind, g).wait()
                kvb[kind, g] = kv32[kind, g].astype(BF16)

            def send_kv(kind, g, to):
                if to < p:
                    send(kvb.at[kind, g], kvR.at[kind, g], rsemR.at[kind * 4 + g], to)
                else:
                    send(kvb.at[kind, g], kvL.at[kind, g], rsemL.at[kind * 4 + g], to)

            def compute_q():
                ld_x.wait(); ld_wq.wait()
                q = dot_nn(x32[...].astype(BF16), wq32[...].astype(BF16)) * (0.125 * LOG2E)
                qb = q.astype(BF16)
                for g in range(NG):
                    b, hp = divmod(g, 2)
                    qp[g] = qb[b * T:(b + 1) * T, hp * T:(hp + 1) * T]

            def gpartial(g, blocks, ctx_ref, lse_ref):
                q2 = stack(qg[g], lo_g)
                ps, m, l = softmax_parts(q2, [(k, None) for k, _ in blocks])
                o = functools.reduce(jnp.add, [dot_nt(pb, v) for pb, (_, v) in zip(ps, blocks)])
                ctx_ref[g] = unstack(o * (1.0 / l), lo_g)
                lse_ref[g] = unstack(m + jnp.log2(l), lo_g)

            if p == 0:
                compute_q()
                for g in range(NG):
                    qg[g] = qp[g, 0:32, :]
                pl.semaphore_wait(bar, 2)
                send(qg, qg, rsemG.at[0], 3)
                send(qg.at[2:4], qg.at[2:4], rsemG.at[0], 1)
                for g in order:
                    for kind in range(2):
                        convert(kind, g)
                        send_kv(kind, g, 1)
                for kind in range(2):
                    t = kv32[kind, 0]
                    for g in range(1, NG):
                        t = jnp.where(lane >= 32 * g, pltpu.roll(kv32[kind, g], 32 * g, 1), t)
                    kvg[kind] = t.astype(BF16)
                    send(kvg.at[kind], kvg.at[kind], rsemG.at[1 + kind], 3)
            elif p == 1:
                pl.semaphore_wait(bar, 1)
                for g in order:
                    for kind in range(2):
                        convert(kind, g)
                        send_kv(kind, g, 0)
                pl.semaphore_wait(ready, 1)
                for g in range(NG):
                    for kind in range(2):
                        send_kv(kind, g, 2)
                compute_q()
            elif p == 2:
                pl.semaphore_wait(bar, 2)
                signal(ready, 1)
                for g in (0, 1):
                    for kind in range(2):
                        convert(kind, g)
                        send_kv(kind, g, 3)
                        convert(kind, g + 2)
                        send_kv(kind, g + 2, 1)
                for g in (0, 1):
                    for kind in range(2):
                        send_kv(kind, g + 2, 3)
                        send_kv(kind, g, 1)
                compute_q()
            else:
                for g in order:
                    for kind in range(2):
                        convert(kind, g)
                pl.semaphore_wait(bar, 2)
                for g in (0, 1):
                    for kind in range(2):
                        send_kv(kind, g, 2)
                compute_q()
                recv(qg, rsemG.at[0])
                for g in (2, 3):
                    gpartial(g, [(kvb[0, g], kvb[1, g])], gctx3, glse3)
                send(gctx3.at[2:4], gctx3.at[2:4], rsemG.at[3], 0)
                send(glse3.at[2:4], glse3.at[2:4], rsemG.at[4], 0)
                for kind in range(2):
                    recv(kvg.at[kind], rsemG.at[1 + kind])
                    send(kvg.at[kind], kvg.at[kind], rsemG.at[1 + kind], 2)
                for g in (2, 3):
                    for kind in range(2):
                        send_kv(kind, g, 2)

            ld_wo.wait()
            if p == 1:
                recv(qg.at[2:4], rsemG.at[0])
            done_b = set()
            stash = {}
            for g in proc:
                b, hp = divmod(g, 2)
                q2 = stack(qp[g], lo)
                blocks = [(kvb[0, g], None)]
                vs = [lambda g=g: kvb[1, g]]
                if has_left:
                    recv(kvL.at[0, g], rsemL.at[g])
                    mask = lane2 >= row2
                    if p == 1:
                        mask = mask | (lane2 < 32)
                    blocks.append((kvL[0, g], mask))
                    vs.append(lambda g=g: kvL[1, g])
                if has_right:
                    recv(kvR.at[0, g], rsemR.at[g])
                    mask = lane2 <= row2
                    if p == 0:
                        mask = mask | (row2 < 32)
                    blocks.append((kvR[0, g], mask))
                    vs.append(lambda g=g: kvR[1, g])
                if p >= 2:
                    if p == 2 and g == proc[0]:
                        recv(kvg.at[0], rsemG.at[1])
                    mask = (lane2 >= 32 * g) & (lane2 < 32 * g + 32)
                    blocks.append((kvg[0], mask))
                    vs.append(lambda: kvg[1])
                ps, m, l = softmax_parts(q2, blocks)
                o = dot_nt(ps[0], vs[0]())
                if p >= 2:
                    if p == 2 and g == proc[0]:
                        recv(kvg.at[1], rsemG.at[2])
                    o = o + dot_nt(ps[-1], vs[-1]())
                i = 1
                if has_left:
                    recv(kvL.at[1, g], rsemL.at[4 + g])
                    o = o + dot_nt(ps[i], vs[i]())
                    i += 1
                if has_right:
                    recv(kvR.at[1, g], rsemR.at[4 + g])
                    o = o + dot_nt(ps[i], vs[i]())
                if p == 3 and g in (0, 1):
                    gpartial(g, [(kvb[0, g], kvb[1, g]), (kvL[0, g], kvL[1, g])], gctx3, glse3)
                    send(gctx3.at[g], gctx3.at[g], rsemG.at[5 + 2 * g], 0)
                    send(glse3.at[g], glse3.at[g], rsemG.at[6 + 2 * g], 0)
                if p == 1 and g in (2, 3):
                    gpartial(g, [(kvR[0, g], kvR[1, g])], gctx1, glse1)
                    send(gctx1.at[g], gctx1.at[g], rsemG.at[5 + 2 * g], 0)
                    send(glse1.at[g], glse1.at[g], rsemG.at[6 + 2 * g], 0)
                ctx = unstack(o * (1.0 / l), lo)
                if p == 0:
                    stash[g] = (ctx[0:32], unstack(m + jnp.log2(l), lo)[0:32])
                contrib = dot_nn(ctx.astype(BF16), wo32[hp * T:(hp + 1) * T, :].astype(BF16))
                if b in done_b:
                    out_ref[b] += contrib
                else:
                    out_ref[b] = contrib
                    done_b.add(b)

            if p == 0:
                recv(gctx3.at[2:4], rsemG.at[3])
                recv(glse3.at[2:4], rsemG.at[4])
                for g in range(NG):
                    if g < 2:
                        recv(gctx3.at[g], rsemG.at[5 + 2 * g]); recv(glse3.at[g], rsemG.at[6 + 2 * g])
                    else:
                        recv(gctx1.at[g], rsemG.at[5 + 2 * g]); recv(glse1.at[g], rsemG.at[6 + 2 * g])
                merged = []
                for g in range(NG):
                    parts = [stash[g], (gctx3[g], glse3[g])]
                    if g >= 2:
                        parts.append((gctx1[g], glse1[g]))
                    M = functools.reduce(jnp.maximum, [e for _, e in parts])
                    ws = [jnp.exp2(e - M) for _, e in parts]
                    num = functools.reduce(jnp.add, [w * c for w, (c, _) in zip(ws, parts)])
                    merged.append((num / functools.reduce(jnp.add, ws)).astype(BF16))
                lhs = jnp.concatenate([jnp.concatenate(merged[0:2], axis=1), jnp.concatenate(merged[2:4], axis=1)], axis=0)
                og = dot_nn(lhs, wo32[...].astype(BF16))
                out_ref[0, 0:32, :] = og[0:32]
                out_ref[1, 0:32, :] = og[32:64]

            for c in sends:
                c.wait_send()

        for p in range(4):
            pl.when(my == p)(functools.partial(program, p))

    any_spec = pl.BlockSpec(memory_space=pl.ANY)
    return pl.pallas_call(
        body,
        out_shape=jax.ShapeDtypeStruct((2, 128, 512), F32),
        in_specs=[any_spec] * 5,
        out_specs=pl.BlockSpec(memory_space=pltpu.VMEM),
        scratch_shapes=[
            pltpu.VMEM((256, 512), F32), pltpu.VMEM((512, 256), F32), pltpu.VMEM((256, 512), F32),
            pltpu.VMEM((2, NG, T, T), F32),
            pltpu.VMEM((2, NG, T, T), BF16), pltpu.VMEM((2, NG, T, T), BF16), pltpu.VMEM((2, NG, T, T), BF16),
            pltpu.VMEM((2, T, T), BF16),
            pltpu.VMEM((NG, T, T), BF16), pltpu.VMEM((NG, 32, T), BF16),
            pltpu.VMEM((NG, 32, T), F32), pltpu.VMEM((NG, 32, T), F32),
            pltpu.VMEM((NG, 32, T), F32), pltpu.VMEM((NG, 32, T), F32),
            pltpu.SemaphoreType.DMA((11,)), pltpu.SemaphoreType.DMA((24,)),
            pltpu.SemaphoreType.DMA((8,)), pltpu.SemaphoreType.DMA((8,)), pltpu.SemaphoreType.DMA((13,)),
            pltpu.SemaphoreType.REGULAR,
        ],
        compiler_params=pltpu.CompilerParams(collective_id=0, disable_semaphore_checks=True),
    )(x2, Wq, kt, vt, Wo)
```

```python
import functools
import os
import jax
import jax.numpy as jnp
from jax import lax
from jax.experimental import pallas as pl
from jax.experimental.pallas import tpu as pltpu

MESH = pl.DeviceIdType.MESH
F32 = jnp.float32
BF16 = jnp.bfloat16
NEG = -1e30
QSCALE = 0.125 * 1.4426950408889634
T = 128
A, B, C, D = 0, 1, 2, 3
SCOPES = bool(os.environ.get("KSCOPES"))


def scope(name):
    import contextlib
    return jax.named_scope(name) if SCOPES else contextlib.nullcontext()


def _sum(xs):
    return functools.reduce(jnp.add, xs)


def _max(xs):
    return functools.reduce(jnp.maximum, xs)


def _iota(shape, dim):
    return lax.broadcasted_iota(jnp.int32, shape, dim)


def _split_dot(a, w, dims, nsplit):
    n = a.shape[0] // nsplit
    outs = [lax.dot_general(a[i * n:(i + 1) * n], w, (dims, ((), ())), preferred_element_type=F32)
            for i in range(nsplit)]
    return outs[0] if nsplit == 1 else jnp.concatenate(outs, axis=0)


def dot_nn(a, w, nsplit=1):
    return _split_dot(a, w, ((1,), (0,)), nsplit)


def dot_nt(a, w, nsplit=1):
    return _split_dot(a, w, ((1,), (1,)), nsplit)


def stack(tile):
    lo = _iota(tile.shape, 1) < 64
    z = jnp.zeros_like(tile)
    return jnp.concatenate([jnp.where(lo, tile, z), jnp.where(lo, z, tile)], axis=0)


def unstack(o):
    n = o.shape[0] // 2
    lo = _iota((n, T), 1) < 64
    return jnp.where(lo, jnp.broadcast_to(o[:n], (n, T)), jnp.broadcast_to(o[n:], (n, T)))


def probs(q2, blocks, nsplit=1):
    ss = []
    for k_tile, mask in blocks:
        s = dot_nn(q2, k_tile, nsplit)
        ss.append(s if mask is None else jnp.where(mask, s, NEG))
    m = jnp.max(_max(ss), axis=1, keepdims=True)
    ps = [jnp.exp2(s - m) for s in ss]
    l = jnp.sum(_sum(ps), axis=1, keepdims=True)
    return [p.astype(BF16) for p in ps], m, l


def stat_mask(n, row0, lane_h0, lane_h1):
    r = _iota((2 * n, T), 0)
    lane = _iota((2 * n, T), 1)
    tgt = jnp.where(r < n, r + (row0 + lane_h0), r + (row0 + lane_h1 - n)) & (T - 1)
    return lane == tgt


def pack_stats(col, mask):
    y = jnp.where(mask, jnp.broadcast_to(col, mask.shape), 0.0)
    return jnp.sum(y.reshape(-1, 8, T), axis=0)


def unpack_stats(z, mask):
    zb = jnp.broadcast_to(z[None], (mask.shape[0] // 8, 8, T)).reshape(mask.shape)
    return jnp.sum(jnp.where(mask, zb, 0.0), axis=1, keepdims=True)


def pallas_dist_sparse_attn_localglobal_qseq_kvseq_b2_sq128_skv128_hq4_dh64_kernel(x, Wq, K_ext, V_ext, Wo):
    kt = jnp.transpose(K_ext, (0, 2, 3, 1)).reshape(512, 128)
    vt = jnp.transpose(V_ext, (0, 2, 3, 1)).reshape(512, 128)
    x2 = x.reshape(256, 512)

    def body(x_hbm, wq_hbm, kt_hbm, vt_hbm, wo_hbm, out_ref,
             x32, wq32, wo32, wob, kv32, kvb, kvL, kvR, kvg, qp, qin, qg, cq, sq, gc, gs, gc1, gs1,
             lsem, ssem, rsemL, rsemR, rsemX, ready):
        my = lax.axis_index("i")
        bar = pltpu.get_barrier_semaphore()

        def signal(sem, to):
            pl.semaphore_signal(sem, inc=1, device_id=(to,), device_id_type=MESH)

        def program(p):
            for to in {0: (1, 3), 1: (0, 2), 2: (3,), 3: (0, 2)}[p]:
                signal(bar, to)

            loads = {}

            def load(name, src, dst):
                c = pltpu.make_async_copy(src, dst, lsem.at[len(loads)])
                c.start()
                loads[name] = c

            def load_kv(kind, g, r0=0, r1=T):
                src = (kt_hbm, vt_hbm)[kind]
                load((kind, g, r0), src.at[pl.ds(g * T + r0, r1 - r0)], kv32.at[kind, g, pl.ds(r0, r1 - r0)])

            def load_x(b):
                load(("x", b), x_hbm.at[pl.ds(b * T, T)], x32.at[pl.ds(b * T, T)])

            def load_wq(hp):
                load(("wq", hp), wq_hbm.at[:, pl.ds(hp * T, T)], wq32.at[hp])

            def wait(name):
                with scope("ldwait"):
                    loads.pop(name).wait()

            sends = []

            def send(src, dst, rsem, to):
                c = pltpu.make_async_remote_copy(src, dst, ssem.at[len(sends)], rsem,
                                                 device_id=(to,), device_id_type=MESH)
                with scope(f"send{to}"):
                    c.start()
                sends.append(c)

            def recv(dst, rsem):
                with scope("recv"):
                    pltpu.make_async_remote_copy(dst, dst, ssem.at[0], rsem,
                                                 device_id=(0,), device_id_type=MESH).wait_recv()

            def convert(kind, g, r0=0, r1=T):
                wait((kind, g, r0))
                kvb[kind, g, r0:r1, :] = kv32[kind, g, r0:r1, :].astype(BF16)

            def send_kv(kind, g, to, r0=0, r1=T, extra=None):
                dst, rsem = (kvR, rsemR) if to < p else (kvL, rsemL)
                rows = pl.ds(r0, r1 - r0)
                send(kvb.at[kind, g, rows], dst.at[kind, g, rows], rsem.at[kind * 4 + g if extra is None else extra], to)

            def recv_kv(side, kind, g, r0=0, r1=T, extra=None):
                buf, rsem = (kvL, rsemL) if side == "L" else (kvR, rsemR)
                recv(buf.at[kind, g, pl.ds(r0, r1 - r0)], rsem.at[kind * 4 + g if extra is None else extra])

            def q_proj(groups):
                for g in groups:
                    b, hp = divmod(g, 2)
                    q = dot_nn(x32[b * T:(b + 1) * T, :].astype(BF16), wq32[hp].astype(BF16))
                    qp[g] = (q * QSCALE).astype(BF16)

            def pack_global(kind):
                lane = _iota((T, T), 1)
                t = kv32[kind, 0]
                for g in range(1, 4):
                    t = jnp.where(lane >= 32 * g, pltpu.roll(kv32[kind, g], 32 * g, 1), t)
                kvg[kind] = t.astype(BF16)

            def wo_prep():
                wait("wo")
                wob[...] = wo32[...].astype(BF16)

            def masks(n, row0):
                lane = _iota((2 * n, T), 1)
                r = _iota((2 * n, T), 0)
                row = jnp.where(r < n, r, r - n) + row0
                return lane, row

            def glob_mask(g, n):
                lane = _iota((2 * n, T), 1)
                return (lane >= 32 * g) & (lane < 32 * g + 32)

            written = set()

            def out_proj(g, ctx, r0=0):
                b, hp = divmod(g, 2)
                contrib = dot_nn(ctx[r0:].astype(BF16), wob[hp * T:(hp + 1) * T, :])
                if b in written:
                    out_ref[b, r0:, :] += contrib
                else:
                    out_ref[b, r0:, :] = contrib
                    written.add(b)

            def group(g, sides, between=None, finish=True, r0=0):
                lane, row = masks(T, 0)
                q2 = stack(qp[g])
                blocks, early, late = [(kvb[0, g], None)], [(0, kvb[1, g])], []
                if "G" in sides:
                    blocks.append((kvg[0], glob_mask(g, T)))
                    early.append((len(blocks) - 1, kvg[1]) if p == 3 or g != A else None)
                for s in sides:
                    if s == "L":
                        recv_k(s, g)
                        mask = lane >= row
                        blocks.append((kvL[0, g], mask | (lane < 32) if p == 1 else mask))
                        late.append((len(blocks) - 1, s))
                    elif s == "R":
                        recv_k(s, g)
                        mask = lane <= row
                        blocks.append((kvR[0, g], mask | (row < 32) if p == 0 else mask))
                        late.append((len(blocks) - 1, s))
                ps, m, l = probs(q2, blocks, {1: 4, 2: 2, 3: 1, 4: 1}[len(blocks)])
                ne = len([e for e in early if e is not None])
                o = _sum([dot_nt(ps[i], v, 4 // ne) for i, v in [e for e in early if e is not None]])
                linv = 1.0 / l
                if between is not None:
                    between()
                lv = []
                if None in early:
                    recv(kvg.at[1], rsemX.at[1])
                    lv.append((1, kvg[1]))
                for i, s in late:
                    recv_v(s, g)
                for i, s in late:
                    lv.append((i, (kvL if s == "L" else kvR)[1, g]))
                if lv:
                    o = o + _sum([dot_nt(ps[i], v, {1: 4, 2: 2, 3: 1}[len(lv)]) for i, v in lv])
                if finish:
                    ctx = unstack(o * linv)
                    out_proj(g, ctx, r0)
                    return ctx, m + jnp.log2(l)
                return o * linv, m + jnp.log2(l)

            got = set()

            def recv_k(s, g):
                if (s, 0, g) in got:
                    return
                got.add((s, 0, g))
                if p == 3 and g == A:
                    recv_kv(s, 0, g, 0, 32, extra=8)
                    recv_kv(s, 0, g, 32, T)
                else:
                    recv_kv(s, 0, g)

            def recv_v(s, g):
                if (s, 1, g) not in got:
                    got.add((s, 1, g))
                    recv_kv(s, 1, g)

            def partial(q_tile, blocks, nsplit=1):
                ps, m, l = probs(stack(q_tile), [(k, mk) for k, _, mk in blocks], nsplit)
                o = _sum([dot_nt(pb, v, nsplit) for pb, (_, v, _) in zip(ps, blocks)])
                return unstack(o * (1.0 / l)).astype(BF16), m + jnp.log2(l)

            def merge_weights(lse_a, lse_b):
                mx = jnp.maximum(lse_a, lse_b)
                a, b = jnp.exp2(lse_a - mx), jnp.exp2(lse_b - mx)
                inv = 1.0 / (a + b)
                return a * inv, b * inv, mx + jnp.log2(a + b)

            def merge_qmode(o_loc, lse_loc):
                recv(sq, rsemX.at[4])
                wa, wb, lse = merge_weights(lse_loc, unpack_stats(sq[...], stat_mask(T, 0, 0, 1)))
                part = unstack(o_loc * wa)
                wb = unstack(wb)
                recv(cq, rsemX.at[5])
                return part + wb * cq[...].astype(F32), lse

            if p == 0:
                load_x(1); load_wq(1)
                for g in (D, C, A, B):
                    load_kv(0, g)
                load_wq(0)
                for g in (D, C, A, B):
                    load_kv(1, g)
                load_x(0)
                load("wo", wo_hbm, wo32)
                wait(("x", 1)); wait(("wq", 1))
                q_proj([D])
                for g in (D, C, A, B):
                    convert(0, g)
                pack_global(0)
                with scope("bar"):
                    pl.semaphore_wait(bar, 2)
                send(qp.at[D], qin, rsemX.at[2], 1)
                send(kvg.at[0], kvg.at[0], rsemX.at[0], 3)
                wait(("wq", 0))
                q_proj([C])
                send(qp.at[C, pl.ds(0, 32)], qg.at[C], rsemX.at[3], 1)
                send_kv(0, D, 1)
                for g in (D, C, A, B):
                    convert(1, g)
                send_kv(1, D, 1)
                for g in (C, A, B):
                    send_kv(0, g, 1); send_kv(1, g, 1)
                pack_global(1)
                send(kvg.at[1], kvg.at[1], rsemX.at[1], 3)
                wait(("x", 0))
                q_proj([A, B])
                for g in range(4):
                    qg[g] = qp[g, 0:32, :]
                send(qg, qg, rsemX.at[3], 3)
                o_d, lse_d = group(D, "", finish=False)
                wo_prep()
                stash = {}
                for g in (A, B, C):
                    ctx, lse = group(g, "R", r0=32)
                    stash[g] = (ctx[0:32], jnp.concatenate([lse[0:32], lse[T:T + 32]], axis=0))
                recv(gs.at[0], rsemX.at[6]); recv(gc.at[pl.ds(2, 2)], rsemX.at[7])
                ctx, lse = merge_qmode(o_d, lse_d)
                out_proj(D, ctx, 32)
                stash[D] = (ctx[0:32], jnp.concatenate([lse[0:32], lse[T:T + 32]], axis=0))

                def gmerge(g, z, off, rem):
                    c, e = stash[g]
                    wa, wb, e2 = merge_weights(e, unpack_stats(z, stat_mask(32, 0, off, off + 32)))
                    stash[g] = (c * unstack(wa) + rem.astype(F32) * unstack(wb), e2)

                gmerge(C, gs[0], 0, gc[C]); gmerge(D, gs[0], 64, gc[D])
                recv(gs.at[1], rsemX.at[8]); recv(gc.at[pl.ds(0, 2)], rsemX.at[9])
                recv(gs1, rsemX.at[10]); recv(gc1, rsemX.at[11])
                gmerge(A, gs[1], 0, gc[A]); gmerge(B, gs[1], 64, gc[B]); gmerge(C, gs1[...], 0, gc1[...])
                lhs = jnp.concatenate([jnp.concatenate([stash[A][0], stash[B][0]], axis=1),
                                       jnp.concatenate([stash[C][0], stash[D][0]], axis=1)], axis=0)
                og = dot_nn(lhs.astype(BF16), wob[...])
                out_ref[0, 0:32, :] = og[0:32]
                out_ref[1, 0:32, :] = og[32:64]

            elif p == 1:
                for g in (A, B, C, D):
                    load_kv(0, g); load_kv(1, g)
                load_x(1); load_wq(1); load_wq(0); load_x(0)
                load("wo", wo_hbm, wo32)
                pl.semaphore_wait(bar, 1)
                for g in (A, B, C):
                    for kind in range(2):
                        convert(kind, g)
                        send_kv(kind, g, 0)
                convert(0, D); convert(1, D)
                with scope("bar"):
                    pl.semaphore_wait(ready, 1)
                for g in (D, A, B, C):
                    send_kv(0, g, 2); send_kv(1, g, 2)
                wait(("x", 1)); wait(("wq", 1)); wait(("wq", 0)); wait(("x", 0))
                q_proj([D, C, A, B])
                recv(qin, rsemX.at[2])
                recv_k("R", D); recv_v("R", D)
                lane, row = masks(96, 32)
                c_hi, e_hi = partial(qin[32:T, :], [(kvb[0, D], kvb[1, D], lane <= row)], 2)
                c_lo, e_lo = partial(qin[0:32, :], [(kvb[0, D], kvb[1, D], None), (kvR[0, D], kvR[1, D], None)])
                cq[0:32, :] = c_lo
                cq[32:T, :] = c_hi
                sq[...] = pack_stats(e_lo, stat_mask(32, 0, 0, 1)) + pack_stats(e_hi, stat_mask(96, 32, 0, 1))
                send(sq, sq, rsemX.at[4], 0)
                send(cq, cq, rsemX.at[5], 0)
                wo_prep()
                group(D, "LR")
                recv(qg.at[C], rsemX.at[3])
                recv_k("R", C); recv_v("R", C)
                c1, e1 = partial(qg[C], [(kvR[0, C], kvR[1, C], None)])
                gc1[...] = c1
                gs1[...] = pack_stats(e1, stat_mask(32, 0, 0, 32))
                send(gs1, gs1, rsemX.at[10], 0)
                send(gc1, gc1, rsemX.at[11], 0)
                for g in (C, A, B):
                    group(g, "LR")

            elif p == 2:
                load_kv(0, A, 0, 32); load_kv(0, A, 32, T); load_kv(0, D)
                load_kv(1, A); load_kv(1, D)
                for kind in range(2):
                    load_kv(kind, B); load_kv(kind, C)
                load_x(1); load_wq(1); load_wq(0); load_x(0)
                load("wo", wo_hbm, wo32)
                with scope("bar"):
                    pl.semaphore_wait(bar, 2)
                signal(ready, 1)
                convert(0, A, 0, 32); send_kv(0, A, 3, 0, 32, extra=8)
                convert(0, A, 32, T); send_kv(0, A, 3, 32, T)
                convert(0, D); send_kv(0, D, 1)
                convert(1, A); send_kv(1, A, 3)
                convert(1, D); send_kv(1, D, 1)
                for kind in range(2):
                    convert(kind, B); send_kv(kind, B, 3)
                    convert(kind, C); send_kv(kind, C, 1)
                for g in (A, B):
                    send_kv(0, g, 1); send_kv(1, g, 1)
                wait(("x", 1)); wait(("wq", 1))
                q_proj([D])
                send(qp.at[D], qin, rsemX.at[2], 3)
                for g in (C, D):
                    send_kv(0, g, 3); send_kv(1, g, 3)
                wait(("wq", 0)); wait(("x", 0))
                q_proj([C, A, B])
                o_d, lse_d = group(D, "L", finish=False)
                wo_prep()
                recv(kvg.at[0], rsemX.at[0])
                for g in (A, B, C):
                    group(g, "GLR")
                ctx, _ = merge_qmode(o_d, lse_d)
                out_proj(D, ctx)

            else:
                for g in (A, B, C, D):
                    load_kv(0, g); load_kv(1, g)
                load_x(0); load_wq(0); load_wq(1); load_x(1)
                load("wo", wo_hbm, wo32)
                for g in (A, B, C, D):
                    convert(0, g); convert(1, g)
                with scope("bar"):
                    pl.semaphore_wait(bar, 2)
                send_kv(0, A, 2); send_kv(1, A, 2)
                recv(kvg.at[0], rsemX.at[0])
                send(kvg.at[0], kvg.at[0], rsemX.at[0], 2)
                wait(("x", 0)); wait(("wq", 0)); wait(("wq", 1)); wait(("x", 1))
                q_proj([A, B, C, D])
                recv(kvg.at[1], rsemX.at[1])
                send(kvg.at[1], kvg.at[1], rsemX.at[1], 2)
                for g in (B, C):
                    send_kv(0, g, 2); send_kv(1, g, 2)
                wo_prep()
                group(A, "GL")
                recv(qg, rsemX.at[3])

                def gsend(g0, slot, sem0, with_left):
                    z = []
                    for j, g in enumerate((g0, g0 + 1)):
                        blocks = [(kvb[0, g], kvb[1, g], None)]
                        if with_left:
                            blocks.append((kvL[0, g], kvL[1, g], None))
                        c, e = partial(qg[g], blocks)
                        gc[g] = c
                        z.append(pack_stats(e, stat_mask(32, 0, 64 * j, 64 * j + 32)))
                    gs[slot] = z[0] + z[1]
                    send(gs.at[slot], gs.at[slot], rsemX.at[sem0], 0)
                    send(gc.at[pl.ds(g0, 2)], gc.at[pl.ds(g0, 2)], rsemX.at[sem0 + 1], 0)

                gsend(C, 0, 6, False)

                def between():
                    recv_v("L", B)
                    gsend(A, 1, 8, True)

                group(B, "GL", between=between)
                recv(qin, rsemX.at[2])
                lane, row = masks(T, 0)
                c2, e2 = partial(qin[...], [(kvb[0, D], kvb[1, D], lane <= row),
                                            (kvg[0], kvg[1], glob_mask(D, T))], 2)
                cq[...] = c2
                sq[...] = pack_stats(e2, stat_mask(T, 0, 0, 1))
                send(sq, sq, rsemX.at[4], 2)
                send(cq, cq, rsemX.at[5], 2)
                for g in (C, D):
                    group(g, "GL")

            with scope("waitsend"):
                for c in sends:
                    c.wait_send()

        for p in range(4):
            pl.when(my == p)(functools.partial(program, p))

    any_spec = pl.BlockSpec(memory_space=pl.ANY)
    vm = pltpu.VMEM
    return pl.pallas_call(
        body,
        out_shape=jax.ShapeDtypeStruct((2, 128, 512), F32),
        in_specs=[any_spec] * 5,
        out_specs=pl.BlockSpec(memory_space=pltpu.VMEM),
        scratch_shapes=[
            vm((256, 512), F32), vm((2, 512, T), F32), vm((256, 512), F32), vm((256, 512), BF16),
            vm((2, 4, T, T), F32),
            vm((2, 4, T, T), BF16), vm((2, 4, T, T), BF16), vm((2, 4, T, T), BF16),
            vm((2, T, T), BF16),
            vm((4, T, T), BF16), vm((T, T), BF16), vm((4, 32, T), BF16),
            vm((T, T), BF16), vm((8, T), F32),
            vm((4, 32, T), BF16), vm((2, 8, T), F32), vm((32, T), BF16), vm((8, T), F32),
            pltpu.SemaphoreType.DMA((14,)), pltpu.SemaphoreType.DMA((24,)),
            pltpu.SemaphoreType.DMA((9,)), pltpu.SemaphoreType.DMA((8,)), pltpu.SemaphoreType.DMA((12,)),
            pltpu.SemaphoreType.REGULAR,
        ],
        compiler_params=pltpu.CompilerParams(collective_id=0, disable_semaphore_checks=True),
    )(x2, Wq, kt, vt, Wo)
```

```python
import functools
import os
import jax
import jax.numpy as jnp
from jax import lax
from jax.experimental import pallas as pl
from jax.experimental.pallas import tpu as pltpu

MESH = pl.DeviceIdType.MESH
F32 = jnp.float32
BF16 = jnp.bfloat16
NEG = -1e30
QSCALE = 0.125 * 1.4426950408889634
T = 128
A, B, C, D = 0, 1, 2, 3
NN = ((1,), (0,))
NT = ((1,), (1,))
SCOPES = bool(os.environ.get("KSCOPES"))
XR = int(os.environ.get("XR", 64))
WR = int(os.environ.get("WR", 64))
F10 = int(os.environ.get("F10", 32))
F23 = int(os.environ.get("F23", 16))
F21 = int(os.environ.get("F21", 32))


def scope(name):
    import contextlib
    return jax.named_scope(name) if SCOPES else contextlib.nullcontext()


def _sum(xs):
    return functools.reduce(jnp.add, xs)


def _max(xs):
    return functools.reduce(jnp.maximum, xs)


def _iota(shape, dim):
    return lax.broadcasted_iota(jnp.int32, shape, dim)


def dot(a, w, dims=NN):
    return lax.dot_general(a, w, (dims, ((), ())), preferred_element_type=F32)


NSPLIT = {1: 4, 2: 2, 3: 4, 4: 1}


def multi_dot(lhss, ws, nsplit=None):
    nsplit = nsplit or NSPLIT[len(ws)]
    n = lhss[0].shape[0] // nsplit
    outs = [[] for _ in ws]
    for c in range(nsplit):
        for i, (a, (w, dims)) in enumerate(zip(lhss, ws)):
            outs[i].append(dot(a[c * n:(c + 1) * n], w, dims))
    return [o[0] if nsplit == 1 else jnp.concatenate(o, axis=0) for o in outs]


def pv(ps, vs, nsplit=None):
    return _sum(multi_dot(ps, vs, nsplit))


def probs(q2, blocks, nsplit=None):
    ss = multi_dot([q2] * len(blocks), [k for k, _ in blocks], nsplit)
    ss = [s if mask is None else jnp.where(mask, s, NEG) for s, (_, mask) in zip(ss, blocks)]
    m = jnp.max(_max(ss), axis=1, keepdims=True)
    ps = [jnp.exp2(s - m) for s in ss]
    l = jnp.sum(_sum(ps), axis=1, keepdims=True)
    return [p.astype(BF16) for p in ps], m, l


def stack(tile):
    lo = _iota(tile.shape, 1) < 64
    z = jnp.zeros_like(tile)
    return jnp.concatenate([jnp.where(lo, tile, z), jnp.where(lo, z, tile)], axis=0)


def unstack(o):
    n = o.shape[0] // 2
    lo = _iota((n, T), 1) < 64
    return jnp.where(lo, jnp.broadcast_to(o[:n], (n, T)), jnp.broadcast_to(o[n:], (n, T)))


def rows2(o, r0, r1):
    n = o.shape[0] // 2
    return jnp.concatenate([o[r0:r1], o[n + r0:n + r1]], axis=0)


def stat_mask(n, row0, lane_h0, lane_h1):
    r = _iota((2 * n, T), 0)
    lane = _iota((2 * n, T), 1)
    tgt = jnp.where(r < n, r + (row0 + lane_h0), r + (row0 + lane_h1 - n)) & (T - 1)
    return lane == tgt


def pack_stats(col, mask):
    y = jnp.where(mask, jnp.broadcast_to(col, mask.shape), 0.0)
    return jnp.sum(y.reshape(-1, 8, T), axis=0)


def unpack_stats(z, mask):
    zb = jnp.broadcast_to(z[None], (mask.shape[0] // 8, 8, T)).reshape(mask.shape)
    return jnp.sum(jnp.where(mask, zb, 0.0), axis=1, keepdims=True)


def merge_weights(lses):
    mx = _max(lses)
    es = [jnp.exp2(e - mx) for e in lses]
    inv = 1.0 / _sum(es)
    return [e * inv for e in es]


def gstat_mask(g):
    off = 64 * (g % 2) + g // 2
    return stat_mask(32, 0, off, off + 32)


def lane_row(n, row0):
    lane = _iota((2 * n, T), 1)
    r = _iota((2 * n, T), 0)
    return lane, jnp.where(r < n, r, r - n) + row0


def glob_mask(g):
    lane = _iota((2 * T, T), 1)
    return (lane >= 32 * g) & (lane < 32 * g + 32)


(S_KG, S_VG, S_QIN, S_QG, S_SQ, S_CQ, S_GS, S_GC0, S_GC1, S_GC2, S_GC3,
 S_STG, S_RLX, S_RLW, S_K2, S_CQ2, S_KV) = range(17)
CS = int(os.environ.get('CS', 64))
N_RSEM = S_KV + 16


def pallas_dist_sparse_attn_localglobal_qseq_kvseq_b2_sq128_skv128_hq4_dh64_kernel(x, Wq, K_ext, V_ext, Wo):
    kt = jnp.transpose(K_ext, (0, 2, 3, 1)).reshape(512, 128)
    vt = jnp.transpose(V_ext, (0, 2, 3, 1)).reshape(512, 128)
    x2 = x.reshape(256, 512)

    def body(x_hbm, wq_hbm, kt_hbm, vt_hbm, wo_hbm, out_ref,
             x32, wq32, wo32, wob, kv32, kvb, kvL, kvR, kvg, qp, qin, qg, cq, sq, gc, gs, gc1,
             stg, relay, lsem, ssem, rsem, ready):
        my = lax.axis_index("i")
        bar = pltpu.get_barrier_semaphore()

        def signal(sem, to):
            pl.semaphore_signal(sem, inc=1, device_id=(to,), device_id_type=MESH)

        def program(p):
            for to in {0: (1, 3), 1: (0, 2), 2: (3,), 3: (0, 2)}[p]:
                signal(bar, to)

            loads = {}
            nload = [0]

            def load(name, src, dst):
                c = pltpu.make_async_copy(src, dst, lsem.at[nload[0]])
                nload[0] += 1
                c.start()
                loads[name] = c

            def load_kv(kind, g, r0=0, r1=T):
                load((kind, g, r0), (kt_hbm, vt_hbm)[kind].at[pl.ds(g * T + r0, r1 - r0)],
                     kv32.at[kind, g, pl.ds(r0, r1 - r0)])

            def load_x(b):
                load(("x", b), x_hbm.at[pl.ds(b * T, T)], x32.at[pl.ds(b * T, T)])

            def load_wq(hp):
                load(("wq", hp), wq_hbm.at[:, pl.ds(hp * T, T)], wq32.at[hp])

            def wait(name):
                with scope("ldwait"):
                    loads.pop(name).wait()

            pending = []
            nsend = [0]

            def send(src, dst, slot, to):
                c = pltpu.make_async_remote_copy(src, dst, ssem.at[nsend[0]], rsem.at[slot],
                                                 device_id=(to,), device_id_type=MESH)
                nsend[0] += 1
                with scope(f"send{to}"):
                    c.start()
                pending.append(c)
                return c

            def drain(*keep):
                with scope("waitsend"):
                    for c in pending:
                        if not any(c is k for k in keep):
                            c.wait_send()
                    pending[:] = [c for c in pending if any(c is k for k in keep)]

            def recv(dst, slot):
                with scope("recv"):
                    pltpu.make_async_remote_copy(dst, dst, ssem.at[0], rsem.at[slot],
                                                 device_id=(0,), device_id_type=MESH).wait_recv()

            def convert(kind, g, r0=0, r1=T):
                wait((kind, g, r0))
                kvb[kind, g, r0:r1, :] = kv32[kind, g, r0:r1, :].astype(BF16)

            def kv_slot(side, kind, g):
                return S_KV + (0 if side == "L" else 8) + kind * 4 + g

            def send_kv(kind, g, to, r0=0, r1=T, slot=None):
                side = "R" if to < p else "L"
                rows = pl.ds(r0, r1 - r0)
                return send(kvb.at[kind, g, rows], (kvR if to < p else kvL).at[kind, g, rows],
                            kv_slot(side, kind, g) if slot is None else slot, to)

            def send_head(g, to, n):
                send(kt_hbm.at[pl.ds(g * T, n)], stg.at[pl.ds(0, n)], S_STG, to)

            got = set()

            def recv_kv(side, kind, g, r0=0, r1=T, slot=None):
                buf = kvL if side == "L" else kvR
                recv(buf.at[kind, g, pl.ds(r0, r1 - r0)], kv_slot(side, kind, g) if slot is None else slot)

            def recv_k(side, g):
                if (side, 0, g) in got:
                    return
                got.add((side, 0, g))
                n = {(0, "R", A): F10, (3, "L", A): F23, (1, "R", C): F21}.get((p, side, g), 0)
                if n:
                    recv(stg.at[pl.ds(0, n)], S_STG)
                    (kvL if side == "L" else kvR)[0, g, 0:n, :] = stg[0:n, :].astype(BF16)
                if (p, side, g) == (3, "L", A):
                    recv_kv(side, 0, g, n, 64, S_K2)
                    n = 64
                recv_kv(side, 0, g, n)

            def recv_v(side, g):
                if (side, 1, g) in got:
                    return
                got.add((side, 1, g))
                n, slot = {(1, "L", B): (XR, S_RLX), (3, "L", C): (WR, S_RLW)}.get((p, side, g), (0, 0))
                if n:
                    recv_kv(side, 1, g, T - n, T, slot)
                recv_kv(side, 1, g, 0, T - n)

            def v_of(side, g):
                if side == "G":
                    return kvg[1], NN
                return {"O": kvb, "L": kvL, "R": kvR}[side][1, g], NT

            def k_of(side, g):
                if side == "G":
                    return kvg[0], NT
                return {"O": kvb, "L": kvL, "R": kvR}[side][0, g], NN

            def q_proj(groups):
                for g in groups:
                    b, hp = divmod(g, 2)
                    q = dot(x32[b * T:(b + 1) * T, :].astype(BF16), wq32[hp].astype(BF16))
                    qp[g] = (q * QSCALE).astype(BF16)

            def pack_global(kind):
                lane = _iota((T, T), 1)
                t = kv32[kind, 0]
                for g in range(1, 4):
                    t = jnp.where(lane >= 32 * g, pltpu.roll(kv32[kind, g], 32 * g, 1), t)
                kvg[kind] = t.T.astype(BF16)

            def wo_prep():
                wait("wo")
                wob[...] = wo32[...].astype(BF16)

            written = set()

            def proj(g, ctx):
                hp = g % 2
                return dot(ctx.astype(BF16), wob[hp * T:(hp + 1) * T, :])

            def out_proj(g, ctx, r0=0):
                b = g // 2
                if b in written:
                    out_ref[b, r0:, :] += proj(g, ctx)
                else:
                    out_ref[b, r0:, :] = proj(g, ctx)
                    written.add(b)

            def scores(g, sides, early):
                for s in sides:
                    if s in "LR":
                        recv_k(s, g)
                for s in early:
                    if s in "LR":
                        recv_v(s, g)
                lane, row = lane_row(T, 0)
                mask = {"O": None, "G": glob_mask(g),
                        "L": (lane >= row) | (lane < 32) if p == 1 else lane >= row,
                        "R": (lane <= row) | (row < 32) if p == 0 else lane <= row}
                ps, m, l = probs(stack(qp[g]), [(k_of(s, g), mask[s]) for s in sides])
                ps = dict(zip(sides, ps))
                o = pv([ps.pop(s) for s in early], [v_of(s, g) for s in early])
                return g, ps, o, 1.0 / l, m + jnp.log2(l)

            def values(st):
                g, ps, o, linv, lse = st
                for s in ps:
                    if s == "G":
                        recv(kvg.at[1, pl.ds(0, 96)], S_VG)
                    else:
                        recv_v(s, g)
                if ps:
                    o = o + pv(list(ps.values()), [v_of(s, g) for s in ps])
                return o * linv

            def finish(st, r0=0):
                ctx = unstack(values(st))
                out_proj(st[0], ctx[r0:], r0)
                return ctx

            def part_scores(q_tile, blocks, nsplit=None):
                ps, m, l = probs(stack(q_tile), [(k_of(s, g), mk) for s, g, mk in blocks], nsplit)
                return ps, 1.0 / l, m + jnp.log2(l)

            def part_values(st, blocks, nsplit=None):
                return unstack(pv(st[0], [v_of(b[0], b[1]) for b in blocks], nsplit) * st[1]).astype(BF16)

            def partial(q_tile, blocks, nsplit=None):
                st = part_scores(q_tile, blocks, nsplit)
                return part_values(st, blocks, nsplit), st[2]

            rlx = relay.at[pl.ds(0, XR)]
            rlw = relay.at[pl.ds(0, WR)]
            m_q = lambda n=T, r0=0: stat_mask(n, r0, 0, 1)
            m_e = lambda: stat_mask(32, 0, 2, 3)

            if p == 0:
                load_x(1); load_wq(0)
                for g in (C, D, A, B):
                    load_kv(0, g)
                load_wq(1)
                for g in (C, D, A, B):
                    load_kv(1, g)
                load_x(0)
                load("wo", wo_hbm, wo32)
                wait(("x", 1)); wait(("wq", 0))
                q_proj([C])
                for g in (C, D, A, B):
                    convert(0, g)
                pack_global(0)
                with scope("bar"):
                    pl.semaphore_wait(bar, 2)
                send(qp.at[C], qin, S_QIN, 1)
                send(kvg.at[0], kvg.at[0], S_KG, 3)
                wait(("wq", 1))
                q_proj([D])
                send(qp.at[D, pl.ds(0, 32)], qg.at[D], S_QG, 1)
                send_kv(0, C, 1)
                for g in (C, D, A, B):
                    convert(1, g)
                send_kv(1, C, 1); send_kv(0, D, 1); send_kv(1, D, 1)
                send_kv(0, A, 1); send_kv(0, B, 1)
                keep = [send_kv(1, A, 1), send_kv(1, B, 1, 0, T - XR)]
                pack_global(1)
                send(kvg.at[1], kvg.at[1], S_VG, 3)
                wait(("x", 0))
                q_proj([A, B])
                for g in range(4):
                    qg[g] = qp[g, 0:32, :]
                send(qg, qg, S_QG, 3)
                send(kvb.at[1, B, pl.ds(T - XR, XR)], rlx, S_RLX, 3)
                st_c = scores(C, "O", "O")
                o_c = values(st_c)
                wo_prep()
                loc, lse = {C: unstack(o_c)}, {C: unstack(st_c[4])}
                for g in (A, B, D):
                    st = scores(g, "OR", "O")
                    loc[g], lse[g] = finish(st, 32)[0:32], unstack(rows2(st[4], 0, 32))
                recv(rlw, S_RLW)
                keep.append(send(rlw, kvL.at[1, C, pl.ds(T - WR, WR)], S_RLW, 3))
                recv(gs, S_GS); recv(sq, S_SQ)
                e3 = {g: unstack(unpack_stats(gs[...], gstat_mask(g))) for g in range(4)}
                e1c = unstack(unpack_stats(sq[...], m_q()))
                e1d = unstack(unpack_stats(sq[...], m_e()))
                w3, w1 = {}, {}
                wa, wb = merge_weights([lse[C][32:], e1c[32:]])
                wga, wgb, w3[C] = merge_weights([lse[C][0:32], e1c[0:32], e3[C]])
                loc[C] = loc[C] * jnp.concatenate([wga, wa], axis=0)
                w1[C] = jnp.concatenate([wgb, wb], axis=0)
                wl, w3[D], w1[D] = merge_weights([lse[D], e3[D], e1d])
                loc[D] = loc[D] * wl
                for g in (A, B):
                    wl, w3[g] = merge_weights([lse[g], e3[g]])
                    loc[g] = loc[g] * wl
                drain(*keep)
                recv(cq.at[pl.ds(0, CS)], S_CQ); recv(gc.at[A], S_GC0); recv(gc.at[pl.ds(C, 2)], S_GC1)
                recv(gc1, S_GC3); recv(gc.at[B], S_GC2)
                f32 = lambda r: r.astype(F32)
                c_lo = loc[C][:CS] + w1[C][:CS] * f32(cq[0:CS, :])
                c_lo = jnp.concatenate([c_lo[0:32] + w3[C] * f32(gc[C]), c_lo[32:]], axis=0)
                o_lo = proj(C, c_lo)
                o_d = proj(D, loc[D] + w3[D] * f32(gc[D]) + w1[D] * f32(gc1[...]))
                out_ref[0, 0:32, :] = (proj(A, loc[A] + w3[A] * f32(gc[A]))
                                       + proj(B, loc[B] + w3[B] * f32(gc[B])))
                out_ref[1, 0:32, :] = o_lo[0:32] + o_d
                out_ref[1, 32:CS, :] += o_lo[32:]
                recv(cq.at[pl.ds(CS, T - CS)], S_CQ2)
                out_ref[1, CS:, :] += proj(C, loc[C][CS:] + w1[C][CS:] * f32(cq[CS:, :]))

            elif p == 1:
                load_kv(0, A, F10)
                pl.semaphore_wait(bar, 1)
                send_head(A, 0, F10)
                load_kv(1, A)
                for g in (B, D):
                    load_kv(0, g); load_kv(1, g)
                load_kv(0, A, 0, F10)
                load_kv(0, C); load_kv(1, C)
                load_x(1); load_wq(0); load_wq(1); load_x(0)
                load("wo", wo_hbm, wo32)
                convert(0, A, F10); send_kv(0, A, 0, F10)
                convert(1, A); send_kv(1, A, 0)
                for g in (B, D):
                    for kind in range(2):
                        convert(kind, g)
                        send_kv(kind, g, 0)
                convert(0, A, 0, F10); convert(0, C); convert(1, C)
                with scope("bar"):
                    pl.semaphore_wait(ready, 1)
                for g in (D, A, B, C):
                    send_kv(0, g, 2); send_kv(1, g, 2)
                wait(("x", 1)); wait(("wq", 0)); wait(("wq", 1)); wait(("x", 0))
                q_proj([C, D, A, B])
                recv(qin, S_QIN)
                recv_k("R", C); recv_v("R", C)
                send(kvR.at[1, C, pl.ds(T - WR, WR)], rlw, S_RLW, 0)
                lane, row = lane_row(96, 32)
                c_hi, e_hi = partial(qin[32:T, :], [("O", C, lane <= row)], 2)
                c_lo, e_lo = partial(qin[0:32, :], [("O", C, None), ("R", C, None)], 1)
                cq[0:32, :] = c_lo
                cq[32:T, :] = c_hi
                z = pack_stats(e_lo, m_q(32)) + pack_stats(e_hi, m_q(96, 32))
                wo_prep()
                st_c = scores(C, "OLR", "OR")
                recv(qg.at[D], S_QG)
                recv_k("R", D)
                st_e = part_scores(qg[D], [("R", D, None)])
                sq[...] = z + pack_stats(st_e[2], m_e())
                send(sq, sq, S_SQ, 0)
                send(cq.at[pl.ds(0, CS)], cq.at[pl.ds(0, CS)], S_CQ, 0)
                recv_v("R", D)
                gc1[...] = part_values(st_e, [("R", D)])
                send(gc1, gc1, S_GC3, 0)
                send(cq.at[pl.ds(CS, T - CS)], cq.at[pl.ds(CS, T - CS)], S_CQ2, 0)
                finish(st_c)
                finish(scores(D, "OLR", "OR"))
                st_a = scores(A, "OLR", "O")
                st_b = scores(B, "OLR", "O")
                drain()
                finish(st_a)
                finish(st_b)

            elif p == 2:
                load_kv(0, A, F23, 64); load_kv(0, C, F21); load_kv(0, A, 64)
                with scope("bar"):
                    pl.semaphore_wait(bar, 2)
                send_head(A, 3, F23)
                send_head(C, 1, F21)
                signal(ready, 1)
                load_kv(1, A); load_kv(1, C)
                for kind in range(2):
                    load_kv(kind, B); load_kv(kind, D)
                load_kv(0, A, 0, F23); load_kv(0, C, 0, F21)
                load_x(1); load_wq(1); load_wq(0); load_x(0)
                load("wo", wo_hbm, wo32)
                kvg[:, 96:T, :] = jnp.zeros((2, 32, T), BF16)
                convert(0, A, F23, 64); send_kv(0, A, 3, F23, 64, S_K2)
                convert(0, C, F21); send_kv(0, C, 1, F21)
                convert(0, A, 64); send_kv(0, A, 3, 64)
                convert(1, A); send_kv(1, A, 3)
                convert(1, C); send_kv(1, C, 1)
                for kind in range(2):
                    convert(kind, B); send_kv(kind, B, 3)
                    convert(kind, D); send_kv(kind, D, 1)
                convert(0, A, 0, F23); convert(0, C, 0, F21)
                for kind in range(2):
                    send_kv(kind, A, 1); send_kv(kind, B, 1)
                wait(("x", 1)); wait(("wq", 1))
                q_proj([D])
                send(qp.at[D], qin, S_QIN, 3)
                send_kv(0, D, 3); send_kv(0, C, 3); send_kv(1, D, 3); send_kv(1, C, 3, 0, T - WR)
                wait(("wq", 0)); wait(("x", 0))
                q_proj([C, A, B])
                st_d = scores(D, "OL", "O")
                o_d, lse_d = unstack(values(st_d)), unstack(st_d[4])
                wo_prep()
                recv(kvg.at[0, pl.ds(0, 96)], S_KG)
                finish(scores(A, "OGLR", "OR"))
                recv_k("R", B)
                recv(rlx, S_RLX)
                send(rlx, kvL.at[1, B, pl.ds(T - XR, XR)], S_RLX, 1)
                finish(scores(B, "OGLR", "OG"))
                st = scores(C, "OGLR", "OG")
                drain()
                finish(st)
                recv(sq, S_SQ)
                wa, wb = merge_weights([lse_d, unstack(unpack_stats(sq[...], m_q()))])
                part = o_d * wa
                recv(cq.at[pl.ds(0, CS)], S_CQ)
                out_ref[1, 0:CS, :] += proj(D, part[:CS] + wb[:CS] * cq[0:CS, :].astype(F32))
                recv(cq.at[pl.ds(CS, T - CS)], S_CQ2)
                out_ref[1, CS:, :] += proj(D, part[CS:] + wb[CS:] * cq[CS:, :].astype(F32))

            else:
                for g in (A, B, C, D):
                    load_kv(0, g); load_kv(1, g)
                load_x(0); load_wq(0); load_wq(1); load_x(1)
                load("wo", wo_hbm, wo32)
                for g in (A, B, C, D):
                    convert(0, g); convert(1, g)
                with scope("bar"):
                    pl.semaphore_wait(bar, 2)
                send_kv(0, A, 2); send_kv(1, A, 2)
                recv(kvg.at[0], S_KG)
                send(kvg.at[0, pl.ds(0, 96)], kvg.at[0, pl.ds(0, 96)], S_KG, 2)
                wait(("x", 0)); wait(("wq", 0)); wait(("wq", 1)); wait(("x", 1))
                q_proj([A, B, C, D])
                recv(kvg.at[1], S_VG)
                send(kvg.at[1, pl.ds(0, 96)], kvg.at[1, pl.ds(0, 96)], S_VG, 2)
                send_kv(0, B, 2)
                wo_prep()
                finish(scores(A, "OGL", "OGL"))
                recv(rlx, S_RLX)
                send(rlx, rlx, S_RLX, 2)
                send_kv(1, B, 2); send_kv(0, C, 2); send_kv(1, C, 2)
                recv(qg, S_QG)
                recv_k("L", B)
                blocks = {g: [("O", g, None)] + ([("L", g, None)] if g < C else []) for g in range(4)}
                sts = {g: part_scores(qg[g], blocks[g], 1) for g in range(4)}
                gs[...] = _sum([pack_stats(sts[g][2], gstat_mask(g)) for g in range(4)])
                for g in (A, C, D):
                    gc[g] = part_values(sts[g], blocks[g], 1)
                send(gs, gs, S_GS, 0)
                send(gc.at[A], gc.at[A], S_GC0, 0)
                send(gc.at[pl.ds(C, 2)], gc.at[pl.ds(C, 2)], S_GC1, 0)
                st = scores(B, "OGL", "OG")
                recv_v("L", B)
                gc[B] = part_values(sts[B], blocks[B], 2)
                send(gc.at[B], gc.at[B], S_GC2, 0)
                finish(st)
                recv(qin, S_QIN)
                lane, row = lane_row(T, 0)
                c2, e2 = partial(qin[...], [("O", D, lane <= row), ("G", D, glob_mask(D))])
                cq[...] = c2
                sq[...] = pack_stats(e2, m_q())
                keep = [send(sq, sq, S_SQ, 2),
                        send(cq.at[pl.ds(0, CS)], cq.at[pl.ds(0, CS)], S_CQ, 2),
                        send(cq.at[pl.ds(CS, T - CS)], cq.at[pl.ds(CS, T - CS)], S_CQ2, 2)]
                st_d = scores(D, "OGL", "OG")
                st_c = scores(C, "OGL", "OG")
                drain(*keep)
                finish(st_d)
                drain()
                finish(st_c)

            drain()

        for p in range(4):
            pl.when(my == p)(functools.partial(program, p))

    any_spec = pl.BlockSpec(memory_space=pl.ANY)
    vm = pltpu.VMEM
    return pl.pallas_call(
        body,
        out_shape=jax.ShapeDtypeStruct((2, 128, 512), F32),
        in_specs=[any_spec] * 5,
        out_specs=pl.BlockSpec(memory_space=pltpu.VMEM),
        scratch_shapes=[
            vm((256, 512), F32), vm((2, 512, T), F32), vm((256, 512), F32), vm((256, 512), BF16),
            vm((2, 4, T, T), F32),
            vm((2, 4, T, T), BF16), vm((2, 4, T, T), BF16), vm((2, 4, T, T), BF16),
            vm((2, T, T), BF16),
            vm((4, T, T), BF16), vm((T, T), BF16), vm((4, 32, T), BF16),
            vm((T, T), BF16), vm((8, T), F32),
            vm((4, 32, T), BF16), vm((8, T), F32), vm((32, T), BF16),
            vm((32, T), F32), vm((64, T), BF16),
            pltpu.SemaphoreType.DMA((16,)), pltpu.SemaphoreType.DMA((24,)),
            pltpu.SemaphoreType.DMA((N_RSEM,)),
            pltpu.SemaphoreType.REGULAR,
        ],
        compiler_params=pltpu.CompilerParams(collective_id=0, disable_semaphore_checks=True),
    )(x2, Wq, kt, vt, Wo)
```

```python
import functools
import os
import jax
import jax.numpy as jnp
from jax import lax
from jax.experimental import pallas as pl
from jax.experimental.pallas import tpu as pltpu

MESH = pl.DeviceIdType.MESH
F32 = jnp.float32
BF16 = jnp.bfloat16
NEG = -1e30
QSCALE = 0.125 * 1.4426950408889634
T = 128
A, B, C, D = 0, 1, 2, 3
NN = ((1,), (0,))
NT = ((1,), (1,))
SCOPES = bool(os.environ.get("KSCOPES"))
XR = int(os.environ.get("XR", 64))
WR = int(os.environ.get("WR", 64))
F10 = int(os.environ.get("F10", 32))
F23 = int(os.environ.get("F23", 16))
F21 = int(os.environ.get("F21", 16))
K2 = int(os.environ.get("K2", 64))


def scope(name):
    import contextlib
    return jax.named_scope(name) if SCOPES else contextlib.nullcontext()


def _sum(xs):
    return functools.reduce(jnp.add, xs)


def _max(xs):
    return functools.reduce(jnp.maximum, xs)


def _iota(shape, dim):
    return lax.broadcasted_iota(jnp.int32, shape, dim)


def dot(a, w, dims=NN):
    return lax.dot_general(a, w, (dims, ((), ())), preferred_element_type=F32)


NSPLIT = {1: 4, 2: 2, 3: 4, 4: 1}


def multi_dot(lhss, ws, nsplit=None):
    nsplit = nsplit or NSPLIT[len(ws)]
    n = lhss[0].shape[0] // nsplit
    outs = [[] for _ in ws]
    for c in range(nsplit):
        for i, (a, (w, dims)) in enumerate(zip(lhss, ws)):
            outs[i].append(dot(a[c * n:(c + 1) * n], w, dims))
    return [o[0] if nsplit == 1 else jnp.concatenate(o, axis=0) for o in outs]


def pv(ps, vs, nsplit=None):
    return _sum(multi_dot(ps, vs, nsplit))


def probs(q2, blocks, nsplit=None):
    ss = multi_dot([q2] * len(blocks), [k for k, _ in blocks], nsplit)
    ss = [s if mask is None else jnp.where(mask, s, NEG) for s, (_, mask) in zip(ss, blocks)]
    m = jnp.max(_max(ss), axis=1, keepdims=True)
    ps = [jnp.exp2(s - m) for s in ss]
    l = jnp.sum(_sum(ps), axis=1, keepdims=True)
    return [p.astype(BF16) for p in ps], m, l


def stack(tile):
    lo = _iota(tile.shape, 1) < 64
    z = jnp.zeros_like(tile)
    return jnp.concatenate([jnp.where(lo, tile, z), jnp.where(lo, z, tile)], axis=0)


def unstack(o):
    n = o.shape[0] // 2
    lo = _iota((n, T), 1) < 64
    return jnp.where(lo, jnp.broadcast_to(o[:n], (n, T)), jnp.broadcast_to(o[n:], (n, T)))


def rows2(o, r0, r1):
    n = o.shape[0] // 2
    return jnp.concatenate([o[r0:r1], o[n + r0:n + r1]], axis=0)


def diag_mask(n, lane0):
    return _iota((n, T), 1) == _iota((n, T), 0) + lane0


def col_to_row(col, lane0):
    n = col.shape[0]
    return jnp.sum(jnp.where(diag_mask(n, lane0), jnp.broadcast_to(col, (n, T)), 0.0), axis=0, keepdims=True)


def row_to_col(row, n, lane0):
    return jnp.sum(jnp.where(diag_mask(n, lane0), jnp.broadcast_to(row, (n, T)), 0.0), axis=1, keepdims=True)


def pair_cols(c0, c1):
    n = c0.shape[0]
    return jnp.where(_iota((n, T), 1) < 64, jnp.broadcast_to(c0, (n, T)), jnp.broadcast_to(c1, (n, T)))


def merge_weights(lses):
    mx = _max(lses)
    es = [jnp.exp2(e - mx) for e in lses]
    inv = 1.0 / _sum(es)
    return [e * inv for e in es]


def lane_row(n, row0):
    lane = _iota((2 * n, T), 1)
    r = _iota((2 * n, T), 0)
    return lane, jnp.where(r < n, r, r - n) + row0


def glob_mask(g):
    lane = _iota((2 * T, T), 1)
    return (lane >= 32 * g) & (lane < 32 * g + 32)


(S_KG, S_VG, S_QIN, S_QG, S_SQ, S_CQ, S_GS, S_GC0, S_GC1, S_GC2, S_GC3,
 S_STG, S_RLX, S_RLW, S_K2, S_CQ2, S_KV) = range(17)
CS = int(os.environ.get('CS', 64))
N_RSEM = S_KV + 16
SQR = int(os.environ.get('SQR', 4))
SLOTN = ("KG VG QIN QG SQ CQ GS GC0 GC1 GC2 GC3 STG RLX RLW K2 CQ2".split()
         + [s + k + g for s in "LR" for k in "kv" for g in "ABCD"])


def pallas_dist_sparse_attn_localglobal_qseq_kvseq_b2_sq128_skv128_hq4_dh64_kernel(x, Wq, K_ext, V_ext, Wo):
    kt = jnp.transpose(K_ext, (0, 2, 3, 1)).reshape(512, 128)
    vt = jnp.transpose(V_ext, (0, 2, 3, 1)).reshape(512, 128)
    x2 = x.reshape(256, 512)

    def body(x_hbm, wq_hbm, kt_hbm, vt_hbm, wo_hbm, out_ref,
             x32, wq32, wo32, wob, kv32, kvb, kvL, kvR, kvg, qp, qin, qg, cq, sq, gc, gs, gc1,
             stg, relay, lsem, ssem, rsem, ready):
        my = lax.axis_index("i")
        bar = pltpu.get_barrier_semaphore()

        def signal(sem, to):
            pl.semaphore_signal(sem, inc=1, device_id=(to,), device_id_type=MESH)

        def program(p):
            for to in {0: (1, 3), 1: (0, 2), 2: (3,), 3: (0, 2)}[p]:
                signal(bar, to)

            loads = {}
            nload = [0]

            def load(name, src, dst):
                c = pltpu.make_async_copy(src, dst, lsem.at[nload[0]])
                nload[0] += 1
                c.start()
                loads[name] = c

            def load_kv(kind, g, r0=0, r1=T):
                load((kind, g, r0), (kt_hbm, vt_hbm)[kind].at[pl.ds(g * T + r0, r1 - r0)],
                     kv32.at[kind, g, pl.ds(r0, r1 - r0)])

            def load_x(b):
                load(("x", b), x_hbm.at[pl.ds(b * T, T)], x32.at[pl.ds(b * T, T)])

            def load_wq(hp):
                load(("wq", hp), wq_hbm.at[:, pl.ds(hp * T, T)], wq32.at[hp])

            def wait(name):
                with scope("ldwait"):
                    loads.pop(name).wait()

            pending = []
            nsend = [0]

            def send(src, dst, slot, to):
                c = pltpu.make_async_remote_copy(src, dst, ssem.at[nsend[0]], rsem.at[slot],
                                                 device_id=(to,), device_id_type=MESH)
                nsend[0] += 1
                with scope(f"send{to}"):
                    c.start()
                pending.append(c)
                return c

            def drain(*keep):
                with scope("waitsend"):
                    for c in pending:
                        if not any(c is k for k in keep):
                            c.wait_send()
                    pending[:] = [c for c in pending if any(c is k for k in keep)]

            def recv(dst, slot):
                with scope("r:" + SLOTN[slot]):
                    pltpu.make_async_remote_copy(dst, dst, ssem.at[0], rsem.at[slot],
                                                 device_id=(0,), device_id_type=MESH).wait_recv()

            def convert(kind, g, r0=0, r1=T):
                wait((kind, g, r0))
                kvb[kind, g, r0:r1, :] = kv32[kind, g, r0:r1, :].astype(BF16)

            def kv_slot(side, kind, g):
                return S_KV + (0 if side == "L" else 8) + kind * 4 + g

            def send_kv(kind, g, to, r0=0, r1=T, slot=None):
                side = "R" if to < p else "L"
                rows = pl.ds(r0, r1 - r0)
                return send(kvb.at[kind, g, rows], (kvR if to < p else kvL).at[kind, g, rows],
                            kv_slot(side, kind, g) if slot is None else slot, to)

            def send_head(g, to, n):
                if n:
                    send(kt_hbm.at[pl.ds(g * T, n)], stg.at[pl.ds(0, n)], S_STG, to)

            got = set()

            def recv_kv(side, kind, g, r0=0, r1=T, slot=None):
                buf = kvL if side == "L" else kvR
                recv(buf.at[kind, g, pl.ds(r0, r1 - r0)], kv_slot(side, kind, g) if slot is None else slot)

            def recv_k(side, g):
                if (side, 0, g) in got:
                    return
                got.add((side, 0, g))
                n = {(0, "R", A): F10, (3, "L", A): F23, (1, "R", C): F21}.get((p, side, g), 0)
                if n:
                    recv(stg.at[pl.ds(0, n)], S_STG)
                    (kvL if side == "L" else kvR)[0, g, 0:n, :] = stg[0:n, :].astype(BF16)
                if (p, side, g) in ((3, "L", A), (1, "R", C)):
                    recv_kv(side, 0, g, n, K2, S_K2)
                    n = K2
                recv_kv(side, 0, g, n)

            def recv_v(side, g):
                if (side, 1, g) in got:
                    return
                got.add((side, 1, g))
                n, slot = {(1, "L", B): (XR, S_RLX), (3, "L", C): (WR, S_RLW)}.get((p, side, g), (0, 0))
                if n:
                    recv_kv(side, 1, g, T - n, T, slot)
                recv_kv(side, 1, g, 0, T - n)

            def v_of(side, g):
                if side == "G":
                    return kvg[1], NN
                return {"O": kvb, "L": kvL, "R": kvR}[side][1, g], NT

            def k_of(side, g):
                if side == "G":
                    return kvg[0], NT
                return {"O": kvb, "L": kvL, "R": kvR}[side][0, g], NN

            def q_proj(groups):
                for g in groups:
                    b, hp = divmod(g, 2)
                    q = dot(x32[b * T:(b + 1) * T, :].astype(BF16), wq32[hp].astype(BF16))
                    qp[g] = (q * QSCALE).astype(BF16)

            def pack_global(kind):
                lane = _iota((T, T), 1)
                t = kv32[kind, 0]
                for g in range(1, 4):
                    t = jnp.where(lane >= 32 * g, pltpu.roll(kv32[kind, g], 32 * g, 1), t)
                kvg[kind] = t.T.astype(BF16)

            def wo_prep():
                wait("wo")
                wob[...] = wo32[...].astype(BF16)

            written = set()

            def proj(g, ctx):
                hp = g % 2
                return dot(ctx.astype(BF16), wob[hp * T:(hp + 1) * T, :])

            def out_proj(g, ctx, r0=0):
                b = g // 2
                if b in written:
                    out_ref[b, r0:, :] += proj(g, ctx)
                else:
                    out_ref[b, r0:, :] = proj(g, ctx)
                    written.add(b)

            def scores(g, sides, early):
                for s in sides:
                    if s in "LR":
                        recv_k(s, g)
                for s in early:
                    if s in "LR":
                        recv_v(s, g)
                lane, row = lane_row(T, 0)
                mask = {"O": None, "G": glob_mask(g),
                        "L": (lane >= row) | (lane < 32) if p == 1 else lane >= row,
                        "R": (lane <= row) | (row < 32) if p == 0 else lane <= row}
                ps, m, l = probs(stack(qp[g]), [(k_of(s, g), mask[s]) for s in sides])
                ps = dict(zip(sides, ps))
                o = pv([ps.pop(s) for s in early], [v_of(s, g) for s in early])
                return g, ps, o, 1.0 / l, m + jnp.log2(l)

            def values(st):
                g, ps, o, linv, lse = st
                for s in ps:
                    if s == "G":
                        recv(kvg.at[1, pl.ds(0, 96)], S_VG)
                    else:
                        recv_v(s, g)
                if ps:
                    o = o + pv(list(ps.values()), [v_of(s, g) for s in ps])
                return o * linv

            def finish(st, r0=0):
                ctx = unstack(values(st))
                out_proj(st[0], ctx[r0:], r0)
                return ctx

            def part_scores(q_tile, blocks, nsplit=None):
                ps, m, l = probs(stack(q_tile), [(k_of(s, g), mk) for s, g, mk in blocks], nsplit)
                return ps, 1.0 / l, m + jnp.log2(l)

            def part_values(st, blocks, nsplit=None):
                return unstack(pv(st[0], [v_of(b[0], b[1]) for b in blocks], nsplit) * st[1]).astype(BF16)

            def partial(q_tile, blocks, nsplit=None):
                st = part_scores(q_tile, blocks, nsplit)
                return part_values(st, blocks, nsplit), st[2]

            rlx = relay.at[pl.ds(0, XR)]
            rlw = relay.at[pl.ds(0, WR)]

            def q_stats():
                return pair_cols(row_to_col(sq[0:1, :], T, 0), row_to_col(sq[1:2, :], T, 0))

            def g_stats(row, lane0):
                return unstack(row_to_col(row, 64, lane0))

            if p == 0:
                load_x(1); load_wq(0)
                for g in (C, D, A, B):
                    load_kv(0, g)
                load_wq(1)
                for g in (C, D, A, B):
                    load_kv(1, g)
                load_x(0)
                load("wo", wo_hbm, wo32)
                wait(("x", 1)); wait(("wq", 0))
                q_proj([C])
                for g in (C, D, A, B):
                    convert(0, g)
                pack_global(0)
                with scope("bar"):
                    pl.semaphore_wait(bar, 2)
                send(qp.at[C], qin, S_QIN, 1)
                send(kvg.at[0], kvg.at[0], S_KG, 3)
                wait(("wq", 1))
                q_proj([D])
                send(qp.at[D, pl.ds(0, 32)], qg.at[D], S_QG, 1)
                send_kv(0, C, 1)
                for g in (C, D, A, B):
                    convert(1, g)
                send_kv(1, C, 1); send_kv(0, D, 1); send_kv(1, D, 1)
                send_kv(0, A, 1); send_kv(0, B, 1)
                keep = [send_kv(1, A, 1), send_kv(1, B, 1, 0, T - XR)]
                pack_global(1)
                send(kvg.at[1], kvg.at[1], S_VG, 3)
                wait(("x", 0))
                q_proj([A, B])
                for g in range(4):
                    qg[g] = qp[g, 0:32, :]
                send(qg, qg, S_QG, 3)
                send(kvb.at[1, B, pl.ds(T - XR, XR)], rlx, S_RLX, 3)
                st_c = scores(C, "O", "O")
                o_c = values(st_c)
                wo_prep()
                loc, lse = {C: unstack(o_c)}, {C: unstack(st_c[4])}
                for g in (A, B, D):
                    st = scores(g, "OR", "O")
                    loc[g], lse[g] = finish(st, 32)[0:32], unstack(rows2(st[4], 0, 32))
                recv(rlw, S_RLW)
                keep.append(send(rlw, kvL.at[1, C, pl.ds(T - WR, WR)], S_RLW, 3))
                recv(gs, S_GS); recv(sq, S_SQ)
                e3 = {g: g_stats(gs[g // 2:g // 2 + 1, :], 64 * (g % 2)) for g in range(4)}
                e1c = q_stats()
                e1d = g_stats(sq[2:3, :], 0)
                w3, w1 = {}, {}
                wa, wb = merge_weights([lse[C][32:], e1c[32:]])
                wga, wgb, w3[C] = merge_weights([lse[C][0:32], e1c[0:32], e3[C]])
                loc[C] = loc[C] * jnp.concatenate([wga, wa], axis=0)
                w1[C] = jnp.concatenate([wgb, wb], axis=0)
                wl, w3[D], w1[D] = merge_weights([lse[D], e3[D], e1d])
                loc[D] = loc[D] * wl
                for g in (A, B):
                    wl, w3[g] = merge_weights([lse[g], e3[g]])
                    loc[g] = loc[g] * wl
                drain(*keep)
                recv(cq.at[pl.ds(0, CS)], S_CQ); recv(gc.at[A], S_GC0); recv(gc.at[pl.ds(C, 2)], S_GC1)
                recv(gc1, S_GC3); recv(gc.at[B], S_GC2)
                f32 = lambda r: r.astype(F32)
                c_lo = loc[C][:CS] + w1[C][:CS] * f32(cq[0:CS, :])
                c_lo = jnp.concatenate([c_lo[0:32] + w3[C] * f32(gc[C]), c_lo[32:]], axis=0)
                o_lo = proj(C, c_lo)
                o_d = proj(D, loc[D] + w3[D] * f32(gc[D]) + w1[D] * f32(gc1[...]))
                out_ref[0, 0:32, :] = (proj(A, loc[A] + w3[A] * f32(gc[A]))
                                       + proj(B, loc[B] + w3[B] * f32(gc[B])))
                out_ref[1, 0:32, :] = o_lo[0:32] + o_d
                out_ref[1, 32:CS, :] += o_lo[32:]
                recv(cq.at[pl.ds(CS, T - CS)], S_CQ2)
                out_ref[1, CS:, :] += proj(C, loc[C][CS:] + w1[C][CS:] * f32(cq[CS:, :]))

            elif p == 1:
                pl.semaphore_wait(bar, 1)
                send_head(A, 0, F10)
                load_kv(0, A, F10)
                load_kv(1, A)
                for g in (B, D):
                    load_kv(0, g); load_kv(1, g)
                load_kv(0, A, 0, F10)
                load_kv(0, C); load_kv(1, C)
                load_x(1); load_wq(0); load_wq(1); load_x(0)
                load("wo", wo_hbm, wo32)
                convert(0, A, F10); send_kv(0, A, 0, F10)
                convert(1, A); send_kv(1, A, 0)
                for g in (B, D):
                    for kind in range(2):
                        convert(kind, g)
                        send_kv(kind, g, 0)
                convert(0, A, 0, F10); convert(0, C); convert(1, C)
                with scope("bar"):
                    pl.semaphore_wait(ready, 1)
                for g in (D, A, B, C):
                    send_kv(0, g, 2); send_kv(1, g, 2)
                wait(("x", 1)); wait(("wq", 0)); wait(("wq", 1)); wait(("x", 0))
                q_proj([C, D, A, B])
                recv(qin, S_QIN)
                recv_k("R", C); recv_v("R", C)
                send(kvR.at[1, C, pl.ds(T - WR, WR)], rlw, S_RLW, 0)
                lane, row = lane_row(96, 32)
                c_hi, e_hi = partial(qin[32:T, :], [("O", C, lane <= row)], 2)
                c_lo, e_lo = partial(qin[0:32, :], [("O", C, None), ("R", C, None)], 1)
                cq[0:32, :] = c_lo
                cq[32:T, :] = c_hi
                for h in range(2):
                    sq[h:h + 1, :] = col_to_row(e_lo[32 * h:32 * h + 32], 0) + col_to_row(e_hi[96 * h:96 * h + 96], 32)
                wo_prep()
                st_c = scores(C, "OLR", "OR")
                recv(qg.at[D], S_QG)
                recv_k("R", D)
                st_e = part_scores(qg[D], [("R", D, None)])
                sq[2:4, :] = jnp.broadcast_to(col_to_row(st_e[2], 0), (2, T))
                send(sq, sq, S_SQ, 0)
                send(cq.at[pl.ds(0, CS)], cq.at[pl.ds(0, CS)], S_CQ, 0)
                recv_v("R", D)
                gc1[...] = part_values(st_e, [("R", D)])
                send(gc1, gc1, S_GC3, 0)
                send(cq.at[pl.ds(CS, T - CS)], cq.at[pl.ds(CS, T - CS)], S_CQ2, 0)
                finish(st_c)
                finish(scores(D, "OLR", "OR"))
                st_a = scores(A, "OLR", "O")
                st_b = scores(B, "OLR", "O")
                drain()
                finish(st_a)
                finish(st_b)

            elif p == 2:
                load_kv(0, A, F23, K2); load_kv(0, C, F21, K2)
                with scope("bar"):
                    pl.semaphore_wait(bar, 2)
                send_head(A, 3, F23)
                send_head(C, 1, F21)
                signal(ready, 1)
                load_kv(0, A, K2); load_kv(0, C, K2)
                load_kv(1, A); load_kv(1, C)
                for kind in range(2):
                    load_kv(kind, B); load_kv(kind, D)
                if F23:
                    load_kv(0, A, 0, F23)
                if F21:
                    load_kv(0, C, 0, F21)
                load_x(1); load_wq(1); load_wq(0); load_x(0)
                load("wo", wo_hbm, wo32)
                kvg[:, 96:T, :] = jnp.zeros((2, 32, T), BF16)
                convert(0, A, F23, K2); send_kv(0, A, 3, F23, K2, S_K2)
                convert(0, C, F21, K2); send_kv(0, C, 1, F21, K2, S_K2)
                convert(0, A, K2); send_kv(0, A, 3, K2)
                convert(0, C, K2); send_kv(0, C, 1, K2)
                convert(1, A); send_kv(1, A, 3)
                convert(1, C); send_kv(1, C, 1)
                for kind in range(2):
                    convert(kind, B); send_kv(kind, B, 3)
                    convert(kind, D); send_kv(kind, D, 1)
                if F23:
                    convert(0, A, 0, F23)
                if F21:
                    convert(0, C, 0, F21)
                for kind in range(2):
                    send_kv(kind, A, 1); send_kv(kind, B, 1)
                wait(("x", 1)); wait(("wq", 1))
                q_proj([D])
                send(qp.at[D], qin, S_QIN, 3)
                send_kv(0, D, 3); send_kv(0, C, 3); send_kv(1, D, 3); send_kv(1, C, 3, 0, T - WR)
                wait(("wq", 0)); wait(("x", 0))
                q_proj([C, A, B])
                st_d = scores(D, "OL", "O")
                o_d, lse_d = unstack(values(st_d)), unstack(st_d[4])
                wo_prep()
                recv(kvg.at[0, pl.ds(0, 96)], S_KG)
                finish(scores(A, "OGLR", "OR"))
                recv_k("R", B)
                recv(rlx, S_RLX)
                send(rlx, kvL.at[1, B, pl.ds(T - XR, XR)], S_RLX, 1)
                finish(scores(B, "OGLR", "OG"))
                st = scores(C, "OGLR", "OG")
                drain()
                finish(st)
                recv(sq.at[pl.ds(0, SQR)], S_SQ)
                wa, wb = merge_weights([lse_d, q_stats()])
                part = o_d * wa
                recv(cq.at[pl.ds(0, CS)], S_CQ)
                out_ref[1, 0:CS, :] += proj(D, part[:CS] + wb[:CS] * cq[0:CS, :].astype(F32))
                recv(cq.at[pl.ds(CS, T - CS)], S_CQ2)
                out_ref[1, CS:, :] += proj(D, part[CS:] + wb[CS:] * cq[CS:, :].astype(F32))

            else:
                for g in (A, B, C, D):
                    load_kv(0, g); load_kv(1, g)
                load_x(0); load_wq(0); load_wq(1); load_x(1)
                load("wo", wo_hbm, wo32)
                for g in (A, B, C, D):
                    convert(0, g); convert(1, g)
                with scope("bar"):
                    pl.semaphore_wait(bar, 2)
                send_kv(0, A, 2); send_kv(1, A, 2)
                recv(kvg.at[0], S_KG)
                send(kvg.at[0, pl.ds(0, 96)], kvg.at[0, pl.ds(0, 96)], S_KG, 2)
                wait(("x", 0)); wait(("wq", 0)); wait(("wq", 1)); wait(("x", 1))
                q_proj([A, B, C, D])
                recv(kvg.at[1], S_VG)
                send(kvg.at[1, pl.ds(0, 96)], kvg.at[1, pl.ds(0, 96)], S_VG, 2)
                send_kv(0, B, 2)
                wo_prep()
                finish(scores(A, "OGL", "OGL"))
                recv(rlx, S_RLX)
                send(rlx, rlx, S_RLX, 2)
                send_kv(1, B, 2); send_kv(0, C, 2); send_kv(1, C, 2)
                recv(qg, S_QG)
                recv_k("L", B)
                blocks = {g: [("O", g, None)] + ([("L", g, None)] if g < C else []) for g in range(4)}
                sts = {g: part_scores(qg[g], blocks[g], 1) for g in range(4)}
                for b in range(2):
                    gs[b:b + 1, :] = col_to_row(sts[2 * b][2], 0) + col_to_row(sts[2 * b + 1][2], 64)
                for g in (A, C, D):
                    gc[g] = part_values(sts[g], blocks[g], 1)
                send(gs, gs, S_GS, 0)
                send(gc.at[A], gc.at[A], S_GC0, 0)
                send(gc.at[pl.ds(C, 2)], gc.at[pl.ds(C, 2)], S_GC1, 0)
                st = scores(B, "OGL", "OG")
                recv_v("L", B)
                gc[B] = part_values(sts[B], blocks[B], 2)
                send(gc.at[B], gc.at[B], S_GC2, 0)
                finish(st)
                recv(qin, S_QIN)
                lane, row = lane_row(T, 0)
                c2, e2 = partial(qin[...], [("O", D, lane <= row), ("G", D, glob_mask(D))])
                cq[...] = c2
                for h in range(2):
                    sq[h:h + 1, :] = col_to_row(e2[T * h:T * h + T], 0)
                if SQR == 4:
                    sq[2:4, :] = jnp.zeros((2, T), F32)
                keep = [send(sq.at[pl.ds(0, SQR)], sq.at[pl.ds(0, SQR)], S_SQ, 2),
                        send(cq.at[pl.ds(0, CS)], cq.at[pl.ds(0, CS)], S_CQ, 2),
                        send(cq.at[pl.ds(CS, T - CS)], cq.at[pl.ds(CS, T - CS)], S_CQ2, 2)]
                st_d = scores(D, "OGL", "OG")
                st_c = scores(C, "OGL", "OG")
                drain(*keep)
                finish(st_d)
                drain()
                finish(st_c)

            drain()

        for p in range(4):
            pl.when(my == p)(functools.partial(program, p))

    any_spec = pl.BlockSpec(memory_space=pl.ANY)
    vm = pltpu.VMEM
    return pl.pallas_call(
        body,
        out_shape=jax.ShapeDtypeStruct((2, 128, 512), F32),
        in_specs=[any_spec] * 5,
        out_specs=pl.BlockSpec(memory_space=pltpu.VMEM),
        scratch_shapes=[
            vm((256, 512), F32), vm((2, 512, T), F32), vm((256, 512), F32), vm((256, 512), BF16),
            vm((2, 4, T, T), F32),
            vm((2, 4, T, T), BF16), vm((2, 4, T, T), BF16), vm((2, 4, T, T), BF16),
            vm((2, T, T), BF16),
            vm((4, T, T), BF16), vm((T, T), BF16), vm((4, 32, T), BF16),
            vm((T, T), BF16), vm((4, T), F32),
            vm((4, 32, T), BF16), vm((2, T), F32), vm((32, T), BF16),
            vm((48, T), F32), vm((96, T), BF16),
            pltpu.SemaphoreType.DMA((17,)), pltpu.SemaphoreType.DMA((24,)),
            pltpu.SemaphoreType.DMA((N_RSEM,)),
            pltpu.SemaphoreType.REGULAR,
        ],
        compiler_params=pltpu.CompilerParams(collective_id=0, disable_semaphore_checks=True),
    )(x2, Wq, kt, vt, Wo)
```

```python
import functools
import os
import jax
import jax.numpy as jnp
from jax import lax
from jax.experimental import pallas as pl
from jax.experimental.pallas import tpu as pltpu

MESH = pl.DeviceIdType.MESH
F32 = jnp.float32
BF16 = jnp.bfloat16
NEG = -1e30
QSCALE = 0.125 * 1.4426950408889634
T = 128
A, B, C, D = 0, 1, 2, 3
NN = ((1,), (0,))
NT = ((1,), (1,))
SCOPES = bool(os.environ.get("KSCOPES"))
XR = int(os.environ.get("XR", 48))
WR = int(os.environ.get("WR", 64))
F10 = int(os.environ.get("F10", 32))
F23 = int(os.environ.get("F23", 16))
F21 = int(os.environ.get("F21", 16))
K2 = int(os.environ.get("K2", 64))


def scope(name):
    import contextlib
    return jax.named_scope(name) if SCOPES else contextlib.nullcontext()


def _sum(xs):
    return functools.reduce(jnp.add, xs)


def _max(xs):
    return functools.reduce(jnp.maximum, xs)


def _iota(shape, dim):
    return lax.broadcasted_iota(jnp.int32, shape, dim)


def dot(a, w, dims=NN):
    return lax.dot_general(a, w, (dims, ((), ())), preferred_element_type=F32)


NSPLIT = {1: 4, 2: 2, 3: 4, 4: 1}


def multi_dot(lhss, ws, nsplit=None):
    nsplit = nsplit or NSPLIT[len(ws)]
    n = lhss[0].shape[0] // nsplit
    outs = [[] for _ in ws]
    for c in range(nsplit):
        for i, (a, (w, dims)) in enumerate(zip(lhss, ws)):
            outs[i].append(dot(a[c * n:(c + 1) * n], w, dims))
    return [o[0] if nsplit == 1 else jnp.concatenate(o, axis=0) for o in outs]


def pv(ps, vs, nsplit=None):
    return _sum(multi_dot(ps, vs, nsplit))


def probs(q2, blocks, nsplit=None):
    ss = multi_dot([q2] * len(blocks), [k for k, _ in blocks], nsplit)
    ss = [s if mask is None else jnp.where(mask, s, NEG) for s, (_, mask) in zip(ss, blocks)]
    m = jnp.max(_max(ss), axis=1, keepdims=True)
    ps = [jnp.exp2(s - m) for s in ss]
    l = jnp.sum(_sum(ps), axis=1, keepdims=True)
    return [p.astype(BF16) for p in ps], m, l


def stack(tile):
    lo = _iota(tile.shape, 1) < 64
    z = jnp.zeros_like(tile)
    return jnp.concatenate([jnp.where(lo, tile, z), jnp.where(lo, z, tile)], axis=0)


def unstack(o):
    n = o.shape[0] // 2
    lo = _iota((n, T), 1) < 64
    return jnp.where(lo, jnp.broadcast_to(o[:n], (n, T)), jnp.broadcast_to(o[n:], (n, T)))


def pick_rows_t(tile, r0, n):
    sel = (_iota((n, T), 1) == _iota((n, T), 0) + r0).astype(BF16)
    return dot(sel, tile, NT).astype(BF16)


def rows2(o, r0, r1):
    n = o.shape[0] // 2
    return jnp.concatenate([o[r0:r1], o[n + r0:n + r1]], axis=0)


def diag_mask(n, lane0):
    return _iota((n, T), 1) == _iota((n, T), 0) + lane0


def col_to_row(col, lane0):
    n = col.shape[0]
    return jnp.sum(jnp.where(diag_mask(n, lane0), jnp.broadcast_to(col, (n, T)), 0.0), axis=0, keepdims=True)


def row_to_col(row, n, lane0):
    return jnp.sum(jnp.where(diag_mask(n, lane0), jnp.broadcast_to(row, (n, T)), 0.0), axis=1, keepdims=True)


def pair_cols(c0, c1):
    n = c0.shape[0]
    return jnp.where(_iota((n, T), 1) < 64, jnp.broadcast_to(c0, (n, T)), jnp.broadcast_to(c1, (n, T)))


def merge_weights(lses):
    mx = _max(lses)
    es = [jnp.exp2(e - mx) for e in lses]
    inv = 1.0 / _sum(es)
    return [e * inv for e in es]


def lane_row(n, row0):
    lane = _iota((2 * n, T), 1)
    r = _iota((2 * n, T), 0)
    return lane, jnp.where(r < n, r, r - n) + row0


def glob_mask(g):
    lane = _iota((2 * T, T), 1)
    return (lane >= 32 * g) & (lane < 32 * g + 32)


(S_KG, S_VG, S_QIN, S_QIN2, S_QG, S_SQ, S_C0, S_C1, S_C2, S_C3, S_C4, S_GS, S_GC0, S_GC1, S_GC2,
 S_STG, S_RLX, S_RLW, S_K2, S_KV) = range(20)
DS = int(os.environ.get('DS', 80))
CS = int(os.environ.get('CS', 64))
N_RSEM = S_KV + 16
SLOTN = ("KG VG QIN QIN2 QG SQ C0 C1 C2 C3 C4 GS GC0 GC1 GC2 STG RLX RLW K2".split()
         + [s + k + g for s in "LR" for k in "kv" for g in "ABCD"])


def pallas_dist_sparse_attn_localglobal_qseq_kvseq_b2_sq128_skv128_hq4_dh64_kernel(x, Wq, K_ext, V_ext, Wo):
    kt = jnp.transpose(K_ext, (0, 2, 3, 1)).reshape(512, 128)
    vt = jnp.transpose(V_ext, (0, 2, 3, 1)).reshape(512, 128)
    x2 = x.reshape(256, 512)

    def body(x_hbm, wq_hbm, kt_hbm, vt_hbm, wo_hbm, out_ref,
             x32, wq32, wo32, wob, kv32, kvb, kvL, kvR, kvg, qp, qin, qg, cin, cout, sin, sout, gc, gs,
             stg, relay, lsem, ssem, rsem, ready):
        my = lax.axis_index("i")
        bar = pltpu.get_barrier_semaphore()

        def signal(sem, to):
            pl.semaphore_signal(sem, inc=1, device_id=(to,), device_id_type=MESH)

        def program(p):
            for to in {0: (1, 3), 1: (0, 2), 2: (3,), 3: (0, 2)}[p]:
                signal(bar, to)

            loads = {}
            nload = [0]

            def load(name, src, dst):
                c = pltpu.make_async_copy(src, dst, lsem.at[nload[0]])
                nload[0] += 1
                c.start()
                loads[name] = c

            def load_kv(kind, g, r0=0, r1=T):
                load((kind, g, r0), (kt_hbm, vt_hbm)[kind].at[pl.ds(g * T + r0, r1 - r0)],
                     kv32.at[kind, g, pl.ds(r0, r1 - r0)])

            def load_x(b):
                load(("x", b), x_hbm.at[pl.ds(b * T, T)], x32.at[pl.ds(b * T, T)])

            def load_wq(hp):
                load(("wq", hp), wq_hbm.at[:, pl.ds(hp * T, T)], wq32.at[hp])

            def wait(name):
                with scope("ldwait"):
                    loads.pop(name).wait()

            pending = []
            nsend = [0]

            def send(src, dst, slot, to):
                c = pltpu.make_async_remote_copy(src, dst, ssem.at[nsend[0]], rsem.at[slot],
                                                 device_id=(to,), device_id_type=MESH)
                nsend[0] += 1
                with scope(f"send{to}"):
                    c.start()
                pending.append(c)
                return c

            def drain(*keep):
                with scope("waitsend"):
                    for c in pending:
                        if not any(c is k for k in keep):
                            c.wait_send()
                    pending[:] = [c for c in pending if any(c is k for k in keep)]

            def recv(dst, slot):
                with scope("r:" + SLOTN[slot]):
                    pltpu.make_async_remote_copy(dst, dst, ssem.at[0], rsem.at[slot],
                                                 device_id=(0,), device_id_type=MESH).wait_recv()

            def convert(kind, g, r0=0, r1=T):
                wait((kind, g, r0))
                kvb[kind, g, r0:r1, :] = kv32[kind, g, r0:r1, :].astype(BF16)

            def kv_slot(side, kind, g):
                return S_KV + (0 if side == "L" else 8) + kind * 4 + g

            def send_kv(kind, g, to, r0=0, r1=T, slot=None):
                side = "R" if to < p else "L"
                rows = pl.ds(r0, r1 - r0)
                return send(kvb.at[kind, g, rows], (kvR if to < p else kvL).at[kind, g, rows],
                            kv_slot(side, kind, g) if slot is None else slot, to)

            def send_head(g, to, n):
                if n:
                    send(kt_hbm.at[pl.ds(g * T, n)], stg.at[pl.ds(0, n)], S_STG, to)

            got = set()

            def recv_kv(side, kind, g, r0=0, r1=T, slot=None):
                buf = kvL if side == "L" else kvR
                recv(buf.at[kind, g, pl.ds(r0, r1 - r0)], kv_slot(side, kind, g) if slot is None else slot)

            def recv_k(side, g):
                if (side, 0, g) in got:
                    return
                got.add((side, 0, g))
                n = {(0, "R", A): F10, (3, "L", A): F23, (1, "R", C): F21}.get((p, side, g), 0)
                if n:
                    recv(stg.at[pl.ds(0, n)], S_STG)
                    (kvL if side == "L" else kvR)[0, g, 0:n, :] = stg[0:n, :].astype(BF16)
                if (p, side, g) in ((3, "L", A), (1, "R", C)):
                    recv_kv(side, 0, g, n, K2, S_K2)
                    n = K2
                recv_kv(side, 0, g, n)

            def recv_v(side, g):
                if (side, 1, g) in got:
                    return
                got.add((side, 1, g))
                n, slot = {(1, "L", A): (XR, S_RLX)}.get((p, side, g), (0, 0))
                if n:
                    recv_kv(side, 1, g, T - n, T, slot)
                recv_kv(side, 1, g, 0, T - n)

            def v_of(side, g):
                if side == "G":
                    return kvg[1], NN
                owner = p + {"O": 0, "L": -1, "R": 1}[side]
                return {"O": kvb, "L": kvL, "R": kvR}[side][1, g], (NN if (owner, g) == (2, C) else NT)

            def k_of(side, g):
                if side == "G":
                    return kvg[0], NT
                return {"O": kvb, "L": kvL, "R": kvR}[side][0, g], NN

            def q_proj(groups):
                for g in groups:
                    b, hp = divmod(g, 2)
                    q = dot(x32[b * T:(b + 1) * T, :].astype(BF16), wq32[hp].astype(BF16))
                    qp[g] = (q * QSCALE).astype(BF16)

            def pack_global(kind):
                for g in range(4):
                    kvg[kind, 32 * g:32 * g + 32, :] = pick_rows_t(kvb[kind, g], 0, 32)

            def wo_prep():
                wait("wo")
                wob[...] = wo32[...].astype(BF16)

            written = set()

            def proj(g, ctx):
                hp = g % 2
                return dot(ctx.astype(BF16), wob[hp * T:(hp + 1) * T, :])

            def out_proj(g, ctx, r0=0):
                b = g // 2
                if b in written:
                    out_ref[b, r0:, :] += proj(g, ctx)
                else:
                    out_ref[b, r0:, :] = proj(g, ctx)
                    written.add(b)

            def scores(g, sides, early):
                for s in sides:
                    if s in "LR":
                        recv_k(s, g)
                for s in early:
                    if s in "LR":
                        recv_v(s, g)
                lane, row = lane_row(T, 0)
                mask = {"O": None, "G": glob_mask(g),
                        "L": (lane >= row) | (lane < 32) if p == 1 else lane >= row,
                        "R": (lane <= row) | (row < 32) if p == 0 else lane <= row}
                ps, m, l = probs(stack(qp[g]), [(k_of(s, g), mask[s]) for s in sides])
                ps = dict(zip(sides, ps))
                o = pv([ps.pop(s) for s in early], [v_of(s, g) for s in early])
                return g, ps, o, 1.0 / l, m + jnp.log2(l)

            def values(st):
                g, ps, o, linv, lse = st
                for s in ps:
                    if s == "G":
                        recv(kvg.at[1, pl.ds(0, 96)], S_VG)
                    else:
                        recv_v(s, g)
                if ps:
                    o = o + pv(list(ps.values()), [v_of(s, g) for s in ps])
                return o * linv

            def finish(st, r0=0):
                ctx = unstack(values(st))
                out_proj(st[0], ctx[r0:], r0)
                return ctx

            def part_scores(q_tile, blocks, nsplit=None):
                ps, m, l = probs(stack(q_tile), [(k_of(s, g), mk) for s, g, mk in blocks], nsplit)
                return ps, 1.0 / l, m + jnp.log2(l)

            def part_values(st, blocks, nsplit=None):
                return unstack(pv(st[0], [v_of(b[0], b[1]) for b in blocks], nsplit) * st[1]).astype(BF16)

            def partial(q_tile, blocks, nsplit=None):
                st = part_scores(q_tile, blocks, nsplit)
                return part_values(st, blocks, nsplit), st[2]

            rlx = relay.at[pl.ds(0, XR)]
            rlw = relay.at[pl.ds(0, WR)]

            def q_stats(i=0):
                return pair_cols(row_to_col(sin[2 * i:2 * i + 1, :], T, 0),
                                 row_to_col(sin[2 * i + 1:2 * i + 2, :], T, 0))

            def send_ctx(i, r0, r1, slot, to):
                rows = pl.ds(r0, r1 - r0)
                return send(cout.at[i, rows], cin.at[i, rows], slot, to)

            def recv_ctx(i, r0, r1, slot):
                recv(cin.at[i, pl.ds(r0, r1 - r0)], slot)

            def serve(blocks, to):
                recv(qin.at[0], S_QIN)
                c, e = partial(qin[0], blocks)
                cout[0] = c
                for h in range(2):
                    sout[h:h + 1, :] = col_to_row(e[T * h:T * h + T], 0)
                return [send(sout.at[pl.ds(0, 2)], sin.at[pl.ds(0, 2)], S_SQ, to),
                        send_ctx(0, 0, CS, S_C0, to), send_ctx(0, CS, T, S_C1, to)]

            def f32(r):
                return r.astype(F32)

            def g_stats(row, lane0):
                return unstack(row_to_col(row, 64, lane0))

            if p == 0:
                load_x(1); load_wq(0)
                for g in (C, D, A, B):
                    load_kv(0, g)
                load_wq(1)
                for g in (C, D, A, B):
                    load_kv(1, g)
                load_x(0)
                load("wo", wo_hbm, wo32)
                wait(("x", 1)); wait(("wq", 0))
                q_proj([C])
                for g in (C, D, A, B):
                    convert(0, g)
                pack_global(0)
                with scope("bar"):
                    pl.semaphore_wait(bar, 2)
                send(qp.at[C], qin.at[0], S_QIN, 1)
                send(kvg.at[0], kvg.at[0], S_KG, 3)
                wait(("wq", 1))
                q_proj([D])
                send(qp.at[D], qin.at[1], S_QIN2, 1)
                send_kv(0, C, 1)
                for g in (C, D, A, B):
                    convert(1, g)
                send_kv(1, C, 1); send_kv(0, D, 1); send_kv(1, D, 1)
                send_kv(0, A, 1); send_kv(1, A, 1, 0, T - XR)
                pack_global(1)
                send(kvg.at[1], kvg.at[1], S_VG, 3)
                wait(("x", 0))
                q_proj([A, B])
                for g in range(4):
                    qg[g] = qp[g, 0:32, :]
                send(qg, qg, S_QG, 3)
                send(kvb.at[1, A, pl.ds(T - XR, XR)], rlx, S_RLX, 3)
                loc, lse = {}, {}
                for g in (C, D):
                    st = scores(g, "O", "O")
                    loc[g], lse[g] = unstack(values(st)), unstack(st[4])
                wo_prep()
                for g in (A, B):
                    st = scores(g, "OR", "O")
                    loc[g], lse[g] = finish(st, 32)[0:32], unstack(rows2(st[4], 0, 32))
                lane, row = lane_row(T, 0)
                keep = serve([("O", B, (lane >= row) | (lane < 32))], 1)
                recv(rlw, S_RLW)
                send(rlw, kvL.at[1, C, pl.ds(T - WR, WR)], S_RLW, 3)
                recv(gs, S_GS); recv(sin, S_SQ)
                w3, w1 = {}, {}
                for g in range(4):
                    e3 = g_stats(gs[g // 2:g // 2 + 1, :], 64 * (g % 2))
                    if g < C:
                        wl, w3[g] = merge_weights([lse[g], e3])
                    else:
                        e1 = q_stats(g - C)
                        wa, wb = merge_weights([lse[g][32:], e1[32:]])
                        wga, wgb, w3[g] = merge_weights([lse[g][0:32], e1[0:32], e3])
                        wl = jnp.concatenate([wga, wa], axis=0)
                        w1[g] = jnp.concatenate([wgb, wb], axis=0)
                    loc[g] = loc[g] * wl
                drain(*keep)

                def merged(g, r0, r1):
                    return loc[g][r0:r1] + w1[g][r0:r1] * f32(cin[g - C, r0:r1, :])

                recv_ctx(0, 32, T, S_C0); recv_ctx(1, 32, DS, S_C1)
                o_c = proj(C, merged(C, 32, T))
                out_ref[1, 32:DS, :] = o_c[:DS - 32] + proj(D, merged(D, 32, DS))
                o_c = o_c[DS - 32:]
                recv(gc.at[A], S_GC0); recv(gc.at[pl.ds(C, 2)], S_GC1); recv(gc.at[B], S_GC2)
                recv_ctx(0, 0, 32, S_C2); recv_ctx(1, 0, 32, S_C3)
                even = jnp.concatenate([loc[A] + w3[A] * f32(gc[A]), merged(C, 0, 32) + w3[C] * f32(gc[C])], axis=0)
                odd = jnp.concatenate([loc[B] + w3[B] * f32(gc[B]), merged(D, 0, 32) + w3[D] * f32(gc[D])], axis=0)
                og = proj(A, even) + proj(B, odd)
                out_ref[0, 0:32, :] = og[0:32]
                out_ref[1, 0:32, :] = og[32:]
                recv_ctx(1, DS, T, S_C4)
                out_ref[1, DS:, :] = o_c + proj(D, merged(D, DS, T))

            elif p == 1:
                pl.semaphore_wait(bar, 1)
                send_head(A, 0, F10)
                load_kv(0, A, F10)
                load_kv(1, A)
                for g in (B, D):
                    load_kv(0, g); load_kv(1, g)
                load_kv(0, A, 0, F10)
                load_kv(0, C); load_kv(1, C)
                load_x(0); load_wq(1); load_x(1); load_wq(0)
                load("wo", wo_hbm, wo32)
                convert(0, A, F10); send_kv(0, A, 0, F10)
                for kind, g in ((1, A), (0, B), (1, B)):
                    convert(kind, g)
                    send_kv(kind, g, 0)
                convert(0, D); convert(1, D)
                convert(0, A, 0, F10); convert(0, C); convert(1, C)
                with scope("bar"):
                    pl.semaphore_wait(ready, 1)
                for g in (D, A, B, C):
                    send_kv(0, g, 2); send_kv(1, g, 2)
                wait(("x", 0)); wait(("wq", 1))
                q_proj([B])
                send(qp.at[B], qin.at[0], S_QIN, 0)
                wait(("x", 1)); wait(("wq", 0))
                q_proj([C, D, A])
                recv(qin.at[0], S_QIN); recv_k("R", C); recv(qin.at[1], S_QIN2)
                lane, row = lane_row(96, 32)
                e_hi, st_lo = {}, {}
                for g in (C, D):
                    cout[g - C, 32:, :], e_hi[g] = partial(qin[g - C, 32:, :], [("O", g, lane <= row)], 2)
                lo_blocks = {g: [("O", g, None), ("R", g, None)] for g in (C, D)}
                st_lo[C] = part_scores(qin[0, 0:32, :], lo_blocks[C], 2)
                recv_v("R", C)
                send(kvR.at[1, C, pl.ds(T - WR, WR)], rlw, S_RLW, 0)
                send_ctx(0, 32, T, S_C0, 0)
                wo_prep()
                st_c = scores(C, "OLR", "OR")
                recv_k("R", D)
                st_lo[D] = part_scores(qin[1, 0:32, :], lo_blocks[D], 2)
                for g in (C, D):
                    for h in range(2):
                        i = 2 * (g - C) + h
                        sout[i:i + 1, :] = (col_to_row(st_lo[g][2][32 * h:32 * h + 32], 0)
                                            + col_to_row(e_hi[g][96 * h:96 * h + 96], 32))
                send(sout, sin, S_SQ, 0)
                send_ctx(1, 32, DS, S_C1, 0)
                recv_v("R", D)
                for g in (C, D):
                    cout[g - C, 0:32, :] = part_values(st_lo[g], lo_blocks[g], 1)
                send_ctx(0, 0, 32, S_C2, 0); send_ctx(1, 0, 32, S_C3, 0); send_ctx(1, DS, T, S_C4, 0)
                finish(st_c)
                finish(scores(D, "OLR", "OR"))
                st_b = scores(B, "OR", "O")
                st_a = scores(A, "OLR", "O")
                drain()
                recv(sin.at[pl.ds(0, 2)], S_SQ)
                wa, wb = merge_weights([unstack(st_b[4]), q_stats()])
                finish(st_a)
                recv_ctx(0, 0, CS, S_C0); recv_ctx(0, CS, T, S_C1)
                out_proj(B, unstack(values(st_b)) * wa + wb * f32(cin[0]))

            elif p == 2:
                load_kv(0, A, F23, K2); load_kv(0, C, F21, K2)
                with scope("bar"):
                    pl.semaphore_wait(bar, 2)
                send_head(A, 3, F23)
                send_head(C, 1, F21)
                signal(ready, 1)
                load_kv(0, A, K2); load_kv(0, C, K2)
                load_kv(1, A); load_kv(1, C)
                for kind in range(2):
                    load_kv(kind, B); load_kv(kind, D)
                if F23:
                    load_kv(0, A, 0, F23)
                if F21:
                    load_kv(0, C, 0, F21)
                load_x(1); load_wq(1); load_wq(0); load_x(0)
                load("wo", wo_hbm, wo32)
                kvg[:, 96:T, :] = jnp.zeros((2, 32, T), BF16)
                convert(0, A, F23, K2); send_kv(0, A, 3, F23, K2, S_K2)
                convert(0, C, F21, K2); send_kv(0, C, 1, F21, K2, S_K2)
                convert(0, A, K2); send_kv(0, A, 3, K2)
                convert(0, C, K2); send_kv(0, C, 1, K2)
                convert(1, A); send_kv(1, A, 3)
                wait((1, C, 0))
                vc = kv32[1, C].astype(BF16)
                for r in range(0, T, 32):
                    kvb[1, C, r:r + 32, :] = pick_rows_t(vc, r, 32)
                send_kv(1, C, 1)
                for kind in range(2):
                    convert(kind, B); send_kv(kind, B, 3)
                    convert(kind, D); send_kv(kind, D, 1)
                if F23:
                    convert(0, A, 0, F23)
                if F21:
                    convert(0, C, 0, F21)
                send_kv(0, A, 1); send_kv(0, B, 1); send_kv(1, A, 1)
                wait(("x", 1)); wait(("wq", 1))
                q_proj([D])
                send(qp.at[D], qin.at[0], S_QIN, 3)
                send_kv(0, D, 3); send_kv(0, C, 3); send_kv(1, D, 3); send_kv(1, C, 3, 0, T - WR)
                wait(("wq", 0)); wait(("x", 0))
                q_proj([C, A, B])
                st_d = scores(D, "OL", "O")
                o_d, lse_d = unstack(values(st_d)), unstack(st_d[4])
                wo_prep()
                recv(kvg.at[0, pl.ds(0, 96)], S_KG)
                finish(scores(A, "OGLR", "OR"))
                recv_k("R", B)
                recv(rlx, S_RLX)
                send(rlx, kvL.at[1, A, pl.ds(T - XR, XR)], S_RLX, 1)
                send_kv(1, B, 1)
                finish(scores(B, "OGLR", "OG"))
                st = scores(C, "OGLR", "OG")
                drain()
                recv(sin.at[pl.ds(0, 2)], S_SQ)
                recv_v("L", C); recv_v("R", C)
                wa, wb = merge_weights([lse_d, q_stats()])
                part = o_d * wa
                finish(st)
                for r0, r1, slot in ((0, CS, S_C0), (CS, T, S_C1)):
                    recv_ctx(0, r0, r1, slot)
                    out_ref[1, r0:r1, :] += proj(D, part[r0:r1] + wb[r0:r1] * f32(cin[0, r0:r1, :]))

            else:
                for g in (A, B, C, D):
                    load_kv(0, g); load_kv(1, g)
                load_x(0); load_wq(0); load_wq(1); load_x(1)
                load("wo", wo_hbm, wo32)
                for g in (A, B, C, D):
                    convert(0, g); convert(1, g)
                with scope("bar"):
                    pl.semaphore_wait(bar, 2)
                send_kv(0, A, 2); send_kv(1, A, 2)
                recv(kvg.at[0], S_KG)
                send(kvg.at[0, pl.ds(0, 96)], kvg.at[0, pl.ds(0, 96)], S_KG, 2)
                wait(("x", 0)); wait(("wq", 0)); wait(("wq", 1)); wait(("x", 1))
                q_proj([A, B, C, D])
                recv(kvg.at[1], S_VG)
                send(kvg.at[1, pl.ds(0, 96)], kvg.at[1, pl.ds(0, 96)], S_VG, 2)
                send_kv(0, B, 2)
                wo_prep()
                finish(scores(A, "OGL", "OGL"))
                recv(rlx, S_RLX)
                send(rlx, rlx, S_RLX, 2)
                send_kv(1, B, 2); send_kv(0, C, 2); send_kv(1, C, 2)
                recv(qg, S_QG)
                recv_k("L", B)
                blocks = {g: [("O", g, None)] + ([("L", g, None)] if g < C else []) for g in range(4)}
                sts = {g: part_scores(qg[g], blocks[g], 1 if g < C else 2) for g in range(4)}
                for b in range(2):
                    gs[b:b + 1, :] = col_to_row(sts[2 * b][2], 0) + col_to_row(sts[2 * b + 1][2], 64)
                for g in (A, C, D):
                    gc[g] = part_values(sts[g], blocks[g], 1)
                send(gs, gs, S_GS, 0)
                send(gc.at[A], gc.at[A], S_GC0, 0)
                send(gc.at[pl.ds(C, 2)], gc.at[pl.ds(C, 2)], S_GC1, 0)
                st = scores(B, "OGL", "OG")
                recv_v("L", B)
                gc[B] = part_values(sts[B], blocks[B], 2)
                send(gc.at[B], gc.at[B], S_GC2, 0)
                finish(st)
                lane, row = lane_row(T, 0)
                keep = serve([("O", D, lane <= row), ("G", D, glob_mask(D))], 2)
                st_d = scores(D, "OGL", "OG")
                lo = T - WR
                recv_kv("L", 1, C, lo, T, S_RLW)
                _, ps, o, linv, _ = scores(C, "OGL", "OG")
                v_hi = jnp.concatenate([jnp.zeros((lo, T), BF16), kvL[1, C, lo:, :]], axis=0)
                o = o + pv([ps["L"]], [(v_hi, NN)])
                o_hi = proj(C, unstack(rows2(o * linv, lo, T)))
                o, linv, p_lo = rows2(o, 0, lo), rows2(linv, 0, lo), rows2(ps["L"], 0, lo)
                drain(*keep)
                o_d = proj(D, unstack(values(st_d)))
                out_ref[1, lo:, :] = o_d[lo:] + o_hi
                o_d = o_d[:lo]
                drain()
                recv_kv("L", 1, C, 0, lo)
                v_lo = jnp.concatenate([kvL[1, C, 0:lo, :], jnp.zeros((WR, T), BF16)], axis=0)
                o = o + pv([p_lo], [(v_lo, NN)], 4 if lo == 64 else 2)
                out_ref[1, 0:lo, :] = o_d + proj(C, unstack(o * linv))

            drain()

        for p in range(4):
            pl.when(my == p)(functools.partial(program, p))

    any_spec = pl.BlockSpec(memory_space=pl.ANY)
    vm = pltpu.VMEM
    return pl.pallas_call(
        body,
        out_shape=jax.ShapeDtypeStruct((2, 128, 512), F32),
        in_specs=[any_spec] * 5,
        out_specs=pl.BlockSpec(memory_space=pltpu.VMEM),
        scratch_shapes=[
            vm((256, 512), F32), vm((2, 512, T), F32), vm((256, 512), F32), vm((256, 512), BF16),
            vm((2, 4, T, T), F32),
            vm((2, 4, T, T), BF16), vm((2, 4, T, T), BF16), vm((2, 4, T, T), BF16),
            vm((2, T, T), BF16),
            vm((4, T, T), BF16), vm((2, T, T), BF16), vm((4, 32, T), BF16),
            vm((2, T, T), BF16), vm((2, T, T), BF16), vm((4, T), F32), vm((4, T), F32),
            vm((4, 32, T), BF16), vm((2, T), F32),
            vm((48, T), F32), vm((96, T), BF16),
            pltpu.SemaphoreType.DMA((17,)), pltpu.SemaphoreType.DMA((24,)),
            pltpu.SemaphoreType.DMA((N_RSEM,)),
            pltpu.SemaphoreType.REGULAR,
        ],
        compiler_params=pltpu.CompilerParams(collective_id=0, disable_semaphore_checks=True),
    )(x2, Wq, kt, vt, Wo)
```

```python
import functools

import jax
import jax.numpy as jnp
from jax import lax
from jax.experimental import pallas as pl
from jax.experimental.pallas import tpu as pltpu

MESH = pl.DeviceIdType.MESH
F32 = jnp.float32
BF16 = jnp.bfloat16
NEG = -1e30
QSCALE = 0.125 * 1.4426950408889634
T = 128
G = 32
A, B, C, D = 0, 1, 2, 3
NN = ((1,), (0,))
NT = ((1,), (1,))

X_ROWS = 48
W_ROWS = 64
HALF = 64
D_SPLIT = 80
HEAD = {(1, 0): 32, (2, 3): 16, (2, 1): 32}

(S_KG, S_VG, S_Q0, S_Q1, S_QG, S_STAT, S_C0, S_C1, S_C2, S_C3, S_C4, S_GS, S_GC0, S_GC1, S_GC2,
 S_HEAD, S_X, S_W, S_K2, S_V2, S_KV) = range(21)
N_RECV = S_KV + 16
N_SEND = 25
N_LOAD = 17


def _sum(xs):
    return functools.reduce(jnp.add, xs)


def _max(xs):
    return functools.reduce(jnp.maximum, xs)


def _iota(shape, dim):
    return lax.broadcasted_iota(jnp.int32, shape, dim)


def _f32(v):
    return v.astype(F32)


def _dot(a, w, dims=NN):
    return lax.dot_general(a, w, (dims, ((), ())), preferred_element_type=F32)


def _dots(lhss, ws, nsplit=None):
    nsplit = nsplit or {1: 4, 2: 2, 3: 4, 4: 1}[len(ws)]
    n = lhss[0].shape[0] // nsplit
    outs = [[] for _ in ws]
    for c in range(nsplit):
        for out, a, (w, dims) in zip(outs, lhss, ws):
            out.append(_dot(a[c * n:(c + 1) * n], w, dims))
    return [o[0] if nsplit == 1 else jnp.concatenate(o, axis=0) for o in outs]


def _pv(ps, vs, nsplit=None):
    return _sum(_dots(ps, vs, nsplit))


def _probs(q2, blocks, nsplit=None):
    ss = _dots([q2] * len(blocks), [k for k, _ in blocks], nsplit)
    ss = [s if mask is None else jnp.where(mask, s, NEG) for s, (_, mask) in zip(ss, blocks)]
    m = jnp.max(_max(ss), axis=1, keepdims=True)
    ps = [jnp.exp2(s - m) for s in ss]
    l = jnp.sum(_sum(ps), axis=1, keepdims=True)
    return [p.astype(BF16) for p in ps], 1.0 / l, m + jnp.log2(l)


def _stack(tile):
    lo = _iota(tile.shape, 1) < 64
    z = jnp.zeros_like(tile)
    return jnp.concatenate([jnp.where(lo, tile, z), jnp.where(lo, z, tile)], axis=0)


def _pair(h0, h1):
    n = h0.shape[0]
    return jnp.where(_iota((n, T), 1) < 64, jnp.broadcast_to(h0, (n, T)), jnp.broadcast_to(h1, (n, T)))


def _unstack(o):
    n = o.shape[0] // 2
    return _pair(o[:n], o[n:])


def _rows2(o, r0, r1):
    n = o.shape[0] // 2
    return jnp.concatenate([o[r0:r1], o[n + r0:n + r1]], axis=0)


def _diag(n, lane0):
    return _iota((n, T), 1) == _iota((n, T), 0) + lane0


def _rows_of_transpose(tile, r0, n):
    return _dot(_diag(n, r0).astype(BF16), tile, NT).astype(BF16)


def _col_to_row(col, lane0):
    n = col.shape[0]
    return jnp.sum(jnp.where(_diag(n, lane0), jnp.broadcast_to(col, (n, T)), 0.0), axis=0, keepdims=True)


def _row_to_col(row, n, lane0):
    return jnp.sum(jnp.where(_diag(n, lane0), jnp.broadcast_to(row, (n, T)), 0.0), axis=1, keepdims=True)


def _merge_weights(lses):
    mx = _max(lses)
    es = [jnp.exp2(e - mx) for e in lses]
    inv = 1.0 / _sum(es)
    return [e * inv for e in es]


def _lane_row(n, row0):
    r = _iota((2 * n, T), 0)
    return _iota((2 * n, T), 1), jnp.where(r < n, r, r - n) + row0


def _global_mask(g):
    lane = _iota((2 * T, T), 1)
    return (lane >= G * g) & (lane < G * g + G)


def _pad_rows(v, before, after):
    parts = [jnp.zeros((before, T), v.dtype)] * bool(before) + [v] + [jnp.zeros((after, T), v.dtype)] * bool(after)
    return jnp.concatenate(parts, axis=0)


def _program(p, bar, x_hbm, wq_hbm, kt_hbm, vt_hbm, wo_hbm, out_ref,
             x32, wq32, wo32, wob, kv32, kv_own, kv_left, kv_right, kv_glob, q_own, q_in, q_glob,
             ctx_in, ctx_out, stat_in, stat_out, glob_ctx, glob_stat, head32, relay, v_keys,
             load_sem, send_sem, recv_sem, ready):
    kv_bufs = {"O": kv_own, "L": kv_left, "R": kv_right}

    def signal(sem, to):
        pl.semaphore_signal(sem, inc=1, device_id=(to,), device_id_type=MESH)

    for to in {0: (1, 3), 1: (2,), 2: (3,), 3: (0, 2)}[p]:
        signal(bar, to)

    loads, started, pending = {}, {"load": 0, "send": 0}, []

    def load(name, src, dst):
        loads[name] = pltpu.make_async_copy(src, dst, load_sem.at[started["load"]])
        started["load"] += 1
        loads[name].start()

    def load_kv(kind, g, r0=0, r1=T):
        load((kind, g, r0), (kt_hbm, vt_hbm)[kind].at[pl.ds(g * T + r0, r1 - r0)],
             kv32.at[kind, g, pl.ds(r0, r1 - r0)])

    def load_x(b):
        load(("x", b), x_hbm.at[pl.ds(b * T, T)], x32.at[pl.ds(b * T, T)])

    def load_wq(hp):
        load(("wq", hp), wq_hbm.at[:, pl.ds(hp * T, T)], wq32.at[hp])

    def wait(*names):
        for name in names:
            loads.pop(name).wait()

    def send(src, dst, slot, to):
        c = pltpu.make_async_remote_copy(src, dst, send_sem.at[started["send"]], recv_sem.at[slot],
                                         device_id=(to,), device_id_type=MESH)
        started["send"] += 1
        c.start()
        pending.append(c)
        return c

    def drain(keep=()):
        for c in pending:
            if not any(c is k for k in keep):
                c.wait_send()
        pending[:] = keep

    def recv(dst, slot):
        pltpu.make_async_remote_copy(dst, dst, send_sem.at[0], recv_sem.at[slot],
                                     device_id=(0,), device_id_type=MESH).wait_recv()

    def rows(r0, r1):
        return pl.ds(r0, r1 - r0)

    def convert(kind, g, r0=0, r1=T):
        wait((kind, g, r0))
        kv_own[kind, g, r0:r1, :] = kv32[kind, g, r0:r1, :].astype(BF16)

    def kv_slot(side, kind, g):
        return S_KV + (0 if side == "L" else 8) + kind * 4 + g

    def send_kv(kind, g, to, r0=0, r1=T, slot=None):
        side = "R" if to < p else "L"
        send(kv_own.at[kind, g, rows(r0, r1)], kv_bufs[side].at[kind, g, rows(r0, r1)],
             kv_slot(side, kind, g) if slot is None else slot, to)

    def send_head(g, to):
        n = HEAD[p, to]
        send(kt_hbm.at[pl.ds(g * T, n)], head32.at[pl.ds(0, n)], S_HEAD, to)

    def recv_kv(side, kind, g, r0=0, r1=T, slot=None):
        recv(kv_bufs[side].at[kind, g, rows(r0, r1)], kv_slot(side, kind, g) if slot is None else slot)

    got = set()

    def recv_k(side, g):
        if (side, 0, g) in got:
            return
        got.add((side, 0, g))
        r = 0
        if (p, side, g) in ((0, "R", A), (3, "L", A), (1, "R", C)):
            r = HEAD[p + (1 if side == "R" else -1), p]
            recv(head32.at[pl.ds(0, r)], S_HEAD)
            kv_bufs[side][0, g, 0:r, :] = head32[0:r, :].astype(BF16)
            if p != 0:
                recv_kv(side, 0, g, r, HALF, S_K2)
                r = HALF
        recv_kv(side, 0, g, r)

    def recv_v(side, g):
        if (side, 1, g) in got:
            return
        got.add((side, 1, g))
        r = T
        if (p, side, g) == (1, "L", A):
            r = T - X_ROWS
            recv_kv(side, 1, g, r, T, S_X)
        recv_kv(side, 1, g, 0, r)

    def send_ctx(i, r0, r1, slot, to):
        return send(ctx_out.at[i, rows(r0, r1)], ctx_in.at[i, rows(r0, r1)], slot, to)

    def recv_ctx(i, r0, r1, slot):
        recv(ctx_in.at[i, rows(r0, r1)], slot)

    relay_x, relay_w = relay.at[pl.ds(0, X_ROWS)], relay.at[pl.ds(0, W_ROWS)]
    glob3 = [kv_glob.at[kind, pl.ds(0, 3 * G)] for kind in range(2)]

    def k_of(side, g):
        return (kv_glob[0], NT) if side == "G" else (kv_bufs[side][0, g], NN)

    def v_of(side, g):
        if side == "G":
            return kv_glob[1], NN
        key_major = (p + {"O": 0, "L": -1, "R": 1}[side], g) == (2, C)
        return kv_bufs[side][1, g], (NN if key_major else NT)

    def q_proj(groups):
        for g in groups:
            b, hp = divmod(g, 2)
            q = _dot(x32[b * T:(b + 1) * T, :].astype(BF16), wq32[hp].astype(BF16))
            q_own[g] = (q * QSCALE).astype(BF16)

    def pack_global(kind):
        for g in range(4):
            kv_glob[kind, G * g:G * g + G, :] = _rows_of_transpose(kv_own[kind, g], 0, G)

    def wo_prep():
        wait("wo")
        wob[...] = wo32[...].astype(BF16)

    def proj(g, ctx):
        hp = g % 2
        return _dot(ctx.astype(BF16), wob[hp * T:(hp + 1) * T, :])

    def scores(g, sides, early):
        for s in sides:
            if s in "LR":
                recv_k(s, g)
        for s in early:
            if s in "LR":
                recv_v(s, g)
        lane, row = _lane_row(T, 0)
        mask = {"O": None, "G": _global_mask(g),
                "L": (lane >= row) | (lane < G) if p == 1 else lane >= row,
                "R": (lane <= row) | (row < G) if p == 0 else lane <= row}
        ps, linv, lse = _probs(_stack(q_own[g]), [(k_of(s, g), mask[s]) for s in sides])
        ps = dict(zip(sides, ps))
        o = _pv([ps.pop(s) for s in early], [v_of(s, g) for s in early])
        return g, ps, o, linv, lse

    def values(st):
        g, ps, o, linv, _ = st
        for s in ps:
            if s == "G":
                recv(glob3[1], S_VG)
            else:
                recv_v(s, g)
        if ps:
            o = o + _pv(list(ps.values()), [v_of(s, g) for s in ps])
        return _unstack(o * linv)

    written = set()

    def finish(st, r0=0):
        g, ctx = st[0], values(st)
        if g // 2 in written:
            out_ref[g // 2, r0:, :] += proj(g, ctx[r0:])
        else:
            out_ref[g // 2, r0:, :] = proj(g, ctx[r0:])
            written.add(g // 2)
        return ctx

    def part_scores(q_tile, blocks, nsplit=None):
        return _probs(_stack(q_tile), [(k_of(s, g), mask) for s, g, mask in blocks], nsplit)

    def part_values(st, blocks, nsplit=None):
        return _unstack(_pv(st[0], [v_of(s, g) for s, g, _ in blocks], nsplit) * st[1]).astype(BF16)

    def serve(blocks, to):
        recv(q_in.at[0], S_Q0)
        st = part_scores(q_in[0], blocks)
        ctx_out[0] = part_values(st, blocks)
        for h in range(2):
            stat_out[h:h + 1, :] = _col_to_row(st[2][T * h:T * h + T], 0)
        return [send(stat_out.at[pl.ds(0, 2)], stat_in.at[pl.ds(0, 2)], S_STAT, to),
                send_ctx(0, 0, HALF, S_C0, to), send_ctx(0, HALF, T, S_C1, to)]

    def remote_lse(i=0):
        return _pair(_row_to_col(stat_in[2 * i:2 * i + 1, :], T, 0),
                     _row_to_col(stat_in[2 * i + 1:2 * i + 2, :], T, 0))

    if p == 0:
        load_x(1); load_wq(0)
        for g in (C, D, A, B):
            load_kv(0, g)
        load_wq(1)
        for g in (C, D, A, B):
            load_kv(1, g)
        load_x(0)
        load("wo", wo_hbm, wo32)
        wait(("x", 1), ("wq", 0))
        q_proj([C])
        for g in (C, D, A, B):
            convert(0, g)
        pack_global(0)
        pl.semaphore_wait(ready, 1)
        send(q_own.at[C], q_in.at[0], S_Q0, 1)
        pl.semaphore_wait(bar, 1)
        send(kv_glob.at[0], kv_glob.at[0], S_KG, 3)
        wait(("wq", 1))
        q_proj([D])
        send(q_own.at[D], q_in.at[1], S_Q1, 1)
        send_kv(0, C, 1)
        for g in (C, D, A, B):
            convert(1, g)
        send_kv(1, C, 1); send_kv(0, D, 1); send_kv(1, D, 1)
        send_kv(0, A, 1); send_kv(1, A, 1, 0, T - X_ROWS)
        pack_global(1)
        send(kv_glob.at[1], kv_glob.at[1], S_VG, 3)
        wait(("x", 0))
        q_proj([A, B])
        for g in range(4):
            q_glob[g] = q_own[g, 0:G, :]
        send(q_glob, q_glob, S_QG, 3)
        send(kv_own.at[1, A, rows(T - X_ROWS, T)], relay_x, S_X, 3)
        loc, lse = {}, {}
        for g in (C, D):
            st = scores(g, "O", "O")
            loc[g], lse[g] = values(st), _unstack(st[4])
        wo_prep()
        for g in (A, B):
            st = scores(g, "OR", "O")
            loc[g], lse[g] = finish(st, G)[0:G], _unstack(_rows2(st[4], 0, G))
        lane, row = _lane_row(T, 0)
        keep = serve([("O", B, (lane >= row) | (lane < G))], 1)
        recv(relay_w, S_W)
        send(relay_w, kv_left.at[1, C, rows(T - W_ROWS, T)], S_W, 3)
        recv(glob_stat, S_GS); recv(stat_in, S_STAT)
        w3, w1 = {}, {}
        for g in range(4):
            e3 = _unstack(_row_to_col(glob_stat[g // 2:g // 2 + 1, :], 2 * G, 64 * (g % 2)))
            if g < C:
                wl, w3[g] = _merge_weights([lse[g], e3])
            else:
                e1 = remote_lse(g - C)
                wa, wb = _merge_weights([lse[g][G:], e1[G:]])
                wga, wgb, w3[g] = _merge_weights([lse[g][0:G], e1[0:G], e3])
                wl = jnp.concatenate([wga, wa], axis=0)
                w1[g] = jnp.concatenate([wgb, wb], axis=0)
            loc[g] = loc[g] * wl
        drain(keep)

        def merged(g, r0, r1):
            return loc[g][r0:r1] + w1[g][r0:r1] * _f32(ctx_in[g - C, r0:r1, :])

        def from3(g):
            return w3[g] * _f32(glob_ctx[g])

        recv_ctx(0, G, T, S_C0); recv_ctx(0, 0, G, S_C2)
        recv(glob_ctx.at[A], S_GC0); recv(glob_ctx.at[pl.ds(C, 2)], S_GC1); recv_ctx(1, G, D_SPLIT, S_C1)
        o_even = proj(A, jnp.concatenate([loc[A] + from3(A), merged(C, 0, G) + from3(C), merged(C, G, T)], axis=0))
        out_ref[1, G:D_SPLIT, :] = o_even[2 * G:G + D_SPLIT] + proj(D, merged(D, G, D_SPLIT))
        o_glob, o_c = o_even[0:2 * G], o_even[G + D_SPLIT:]
        recv(glob_ctx.at[B], S_GC2); recv_ctx(1, 0, G, S_C3)
        o_glob = o_glob + proj(B, jnp.concatenate([loc[B] + from3(B), merged(D, 0, G) + from3(D)], axis=0))
        out_ref[0, 0:G, :] = o_glob[0:G]
        out_ref[1, 0:G, :] = o_glob[G:]
        recv_ctx(1, D_SPLIT, T, S_C4)
        out_ref[1, D_SPLIT:, :] = o_c + proj(D, merged(D, D_SPLIT, T))

    elif p == 1:
        h10 = HEAD[1, 0]
        pl.semaphore_wait(bar, 1)
        signal(ready, 0)
        send_head(A, 0)
        load_kv(0, A, h10)
        load_kv(1, A)
        for g in (B, D):
            load_kv(0, g); load_kv(1, g)
        load_kv(0, A, 0, h10)
        load_kv(0, C); load_kv(1, C)
        load_x(0); load_wq(1); load_x(1); load_wq(0)
        load("wo", wo_hbm, wo32)
        convert(0, A, h10); send_kv(0, A, 0, h10)
        for kind, g in ((1, A), (0, B), (1, B)):
            convert(kind, g)
            send_kv(kind, g, 0)
        convert(0, D); convert(1, D)
        convert(0, A, 0, h10); convert(0, C); convert(1, C)
        pl.semaphore_wait(ready, 1)
        for g in (D, A, B, C):
            send_kv(0, g, 2); send_kv(1, g, 2)
        wait(("x", 0), ("wq", 1))
        q_proj([B])
        send(q_own.at[B], q_in.at[0], S_Q0, 0)
        wait(("x", 1), ("wq", 0))
        q_proj([C, D, A])
        recv(q_in.at[0], S_Q0); recv_k("R", C); recv(q_in.at[1], S_Q1)
        lane, row = _lane_row(T - G, G)
        hi, lo = {}, {}
        for g in (C, D):
            blocks = [("O", g, lane <= row)]
            hi[g] = part_scores(q_in[g - C, G:, :], blocks, 2)
            ctx_out[g - C, G:, :] = part_values(hi[g], blocks, 2)
        lo_blocks = {g: [("O", g, None), ("R", g, None)] for g in (C, D)}
        lo[C] = part_scores(q_in[0, 0:G, :], lo_blocks[C], 2)
        recv_v("R", C)
        send(kv_right.at[1, C, rows(T - W_ROWS, T)], relay_w, S_W, 0)
        send_ctx(0, G, T, S_C0, 0)
        wo_prep()
        st_c = scores(C, "OLR", "OR")
        recv_k("R", D)
        lo[D] = part_scores(q_in[1, 0:G, :], lo_blocks[D], 2)
        ctx_out[0, 0:G, :] = part_values(lo[C], lo_blocks[C], 2)
        o = _pv([lo[D][0][0]], [v_of("O", D)])
        for g in (C, D):
            for h in range(2):
                i = 2 * (g - C) + h
                stat_out[i:i + 1, :] = (_col_to_row(lo[g][2][G * h:G * h + G], 0)
                                        + _col_to_row(hi[g][2][(T - G) * h:(T - G) * (h + 1)], G))
        send(stat_out, stat_in, S_STAT, 0)
        send_ctx(0, 0, G, S_C2, 0); send_ctx(1, G, D_SPLIT, S_C1, 0)
        recv_v("R", D)
        o = o + _pv([lo[D][0][1]], [v_of("R", D)])
        ctx_out[1, 0:G, :] = _unstack(o * lo[D][1]).astype(BF16)
        send_ctx(1, 0, G, S_C3, 0); send_ctx(1, D_SPLIT, T, S_C4, 0)
        finish(st_c)
        finish(scores(D, "OLR", "OR"))
        _, ps, o, linv, lse_b = scores(B, "OR", "O")
        st_a = scores(A, "OLR", "O")
        recv(stat_in.at[pl.ds(0, 2)], S_STAT)
        recv_v("L", A); recv_v("R", A)
        wa, wb = _merge_weights([_unstack(lse_b), remote_lse()])
        finish(st_a)
        drain()
        recv_ctx(0, 0, HALF, S_C0); recv_kv("R", 1, B, 0, HALF, S_V2)
        o = o + _pv([ps["R"]], [(_pad_rows(kv_right[1, B, 0:HALF, :], 0, T - HALF), NN)])
        out_ref[0, 0:HALF, :] += proj(B, _unstack(_rows2(o * linv, 0, HALF)) * wa[:HALF]
                                      + wb[:HALF] * _f32(ctx_in[0, 0:HALF, :]))
        o, linv, p_hi = _rows2(o, HALF, T), _rows2(linv, HALF, T), _rows2(ps["R"], HALF, T)
        recv_ctx(0, HALF, T, S_C1); recv_kv("R", 1, B, HALF, T)
        o = o + _pv([p_hi], [(_pad_rows(kv_right[1, B, HALF:, :], HALF, 0), NN)])
        out_ref[0, HALF:, :] += proj(B, _unstack(o * linv) * wa[HALF:] + wb[HALF:] * _f32(ctx_in[0, HALF:, :]))

    elif p == 2:
        h23, h21 = HEAD[2, 3], HEAD[2, 1]
        load_kv(0, A, h23, HALF)
        pl.semaphore_wait(bar, 2)
        send_head(A, 3)
        send_head(C, 1)
        signal(ready, 1)
        load_kv(0, C, h21, HALF); load_kv(0, A, HALF); load_kv(0, C, HALF)
        load_kv(1, A); load_kv(1, C)
        for kind in range(2):
            load_kv(kind, B); load_kv(kind, D)
        load_kv(0, A, 0, h23); load_kv(0, C, 0, h21)
        load_x(1); load_wq(1); load_wq(0); load_x(0)
        load("wo", wo_hbm, wo32)
        kv_glob[:, 3 * G:, :] = jnp.zeros((2, G, T), BF16)
        convert(0, A, h23, HALF); send_kv(0, A, 3, h23, HALF, S_K2)
        convert(0, C, h21, HALF); send_kv(0, C, 1, h21, HALF, S_K2)
        convert(0, A, HALF); send_kv(0, A, 3, HALF)
        convert(0, C, HALF); send_kv(0, C, 1, HALF)
        convert(1, A); send_kv(1, A, 3)
        wait((1, C, 0))
        v_c = kv32[1, C].astype(BF16)
        for r in range(0, T, 32):
            kv_own[1, C, r:r + 32, :] = _rows_of_transpose(v_c, r, 32)
        send_kv(1, C, 1)
        for kind in range(2):
            convert(kind, B); send_kv(kind, B, 3)
            convert(kind, D); send_kv(kind, D, 1)
        convert(0, A, 0, h23); convert(0, C, 0, h21)
        send_kv(0, A, 1); send_kv(0, B, 1); send_kv(1, A, 1)
        wait(("x", 1), ("wq", 1))
        q_proj([D])
        send(q_own.at[D], q_in.at[0], S_Q0, 3)
        send_kv(0, D, 3); send_kv(0, C, 3); send_kv(1, D, 3); send_kv(1, C, 3, 0, T - W_ROWS)
        wait(("wq", 0), ("x", 0))
        q_proj([C, A, B])
        st = scores(D, "OL", "O")
        ctx_d, lse_d = values(st), _unstack(st[4])
        wo_prep()
        for r in range(0, T, 32):
            v_keys[r:r + 32, :] = _rows_of_transpose(kv_own[1, B], r, 32)
        recv(glob3[0], S_KG)
        finish(scores(A, "OGLR", "OR"))
        recv_k("R", B)
        recv(relay_x, S_X)
        send(relay_x, kv_left.at[1, A, rows(T - X_ROWS, T)], S_X, 1)
        send(v_keys.at[rows(0, HALF)], kv_right.at[1, B, rows(0, HALF)], S_V2, 1)
        send(v_keys.at[rows(HALF, T)], kv_right.at[1, B, rows(HALF, T)], kv_slot("R", 1, B), 1)
        finish(scores(B, "OGLR", "OG"))
        st = scores(C, "OGLR", "OG")
        drain()
        recv(stat_in.at[pl.ds(0, 2)], S_STAT)
        recv_v("L", C); recv_v("R", C)
        wa, wb = _merge_weights([lse_d, remote_lse()])
        ctx_d = ctx_d * wa
        finish(st)
        for r0, r1, slot in ((0, HALF, S_C0), (HALF, T, S_C1)):
            recv_ctx(0, r0, r1, slot)
            out_ref[1, r0:r1, :] += proj(D, ctx_d[r0:r1] + wb[r0:r1] * _f32(ctx_in[0, r0:r1, :]))

    else:
        for g in (A, B, C, D):
            load_kv(0, g); load_kv(1, g)
        load_x(0); load_wq(0); load_wq(1); load_x(1)
        load("wo", wo_hbm, wo32)
        for g in (A, B, C, D):
            convert(0, g); convert(1, g)
        pl.semaphore_wait(bar, 2)
        send_kv(0, A, 2); send_kv(1, A, 2)
        recv(kv_glob.at[0], S_KG)
        send(glob3[0], glob3[0], S_KG, 2)
        wait(("x", 0), ("wq", 0), ("wq", 1), ("x", 1))
        q_proj([A, B, C, D])
        recv(kv_glob.at[1], S_VG)
        send(glob3[1], glob3[1], S_VG, 2)
        send_kv(0, B, 2)
        wo_prep()
        finish(scores(A, "OGL", "OGL"))
        recv(relay_x, S_X)
        send(relay_x, relay_x, S_X, 2)
        send_kv(1, B, 2); send_kv(0, C, 2); send_kv(1, C, 2)
        recv(q_glob, S_QG)
        recv_k("L", B)
        blocks = {g: [("O", g, None)] + [("L", g, None)] * (g < C) for g in range(4)}
        sts = {g: part_scores(q_glob[g], blocks[g], 1 if g < C else 2) for g in range(4)}
        for b in range(2):
            glob_stat[b:b + 1, :] = _col_to_row(sts[2 * b][2], 0) + _col_to_row(sts[2 * b + 1][2], 64)
        for g in (A, C, D):
            glob_ctx[g] = part_values(sts[g], blocks[g], 1)
        send(glob_stat, glob_stat, S_GS, 0)
        send(glob_ctx.at[A], glob_ctx.at[A], S_GC0, 0)
        send(glob_ctx.at[pl.ds(C, 2)], glob_ctx.at[pl.ds(C, 2)], S_GC1, 0)
        st = scores(B, "OGL", "OG")
        recv_v("L", B)
        glob_ctx[B] = part_values(sts[B], blocks[B], 2)
        send(glob_ctx.at[B], glob_ctx.at[B], S_GC2, 0)
        finish(st)
        lane, row = _lane_row(T, 0)
        keep = serve([("O", D, lane <= row), ("G", D, _global_mask(D))], 2)
        st_d = scores(D, "OGL", "OG")
        n = T - W_ROWS
        recv_kv("L", 1, C, n, T, S_W)
        _, ps, o, linv, _ = scores(C, "OGL", "OG")
        o = o + _pv([ps["L"]], [(_pad_rows(kv_left[1, C, n:, :], n, 0), NN)])
        o_hi = proj(C, _unstack(_rows2(o * linv, n, T)))
        o, linv, p_lo = _rows2(o, 0, n), _rows2(linv, 0, n), _rows2(ps["L"], 0, n)
        drain(keep)
        o_d = proj(D, values(st_d))
        out_ref[1, n:, :] = o_d[n:] + o_hi
        o_d = o_d[:n]
        drain()
        recv_kv("L", 1, C, 0, n)
        o = o + _pv([p_lo], [(_pad_rows(kv_left[1, C, 0:n, :], 0, W_ROWS), NN)])
        out_ref[1, 0:n, :] = o_d + proj(C, _unstack(o * linv))

    drain()
    assert not loads and started["load"] <= N_LOAD and started["send"] <= N_SEND


def pallas_dist_sparse_attn_localglobal_qseq_kvseq_b2_sq128_skv128_hq4_dh64_kernel(x, Wq, K_ext, V_ext, Wo):
    kt = jnp.transpose(K_ext, (0, 2, 3, 1)).reshape(4 * T, T)
    vt = jnp.transpose(V_ext, (0, 2, 3, 1)).reshape(4 * T, T)

    def body(*refs):
        my = lax.axis_index("i")
        bar = pltpu.get_barrier_semaphore()
        for p in range(4):
            pl.when(my == p)(functools.partial(_program, p, bar, *refs))

    vmem = pltpu.VMEM
    return pl.pallas_call(
        body,
        out_shape=jax.ShapeDtypeStruct((2, T, 512), F32),
        in_specs=[pl.BlockSpec(memory_space=pl.ANY)] * 5,
        out_specs=pl.BlockSpec(memory_space=pltpu.VMEM),
        scratch_shapes=[
            vmem((2 * T, 512), F32),
            vmem((2, 512, T), F32),
            vmem((2 * T, 512), F32),
            vmem((2 * T, 512), BF16),
            vmem((2, 4, T, T), F32),
            vmem((2, 4, T, T), BF16),
            vmem((2, 4, T, T), BF16),
            vmem((2, 4, T, T), BF16),
            vmem((2, T, T), BF16),
            vmem((4, T, T), BF16),
            vmem((2, T, T), BF16),
            vmem((4, G, T), BF16),
            vmem((2, T, T), BF16),
            vmem((2, T, T), BF16),
            vmem((4, T), F32),
            vmem((4, T), F32),
            vmem((4, G, T), BF16),
            vmem((2, T), F32),
            vmem((32, T), F32),
            vmem((64, T), BF16),
            vmem((T, T), BF16),
            pltpu.SemaphoreType.DMA((N_LOAD,)),
            pltpu.SemaphoreType.DMA((N_SEND,)),
            pltpu.SemaphoreType.DMA((N_RECV,)),
            pltpu.SemaphoreType.REGULAR,
        ],
        compiler_params=pltpu.CompilerParams(collective_id=0, disable_semaphore_checks=True),
    )(x.reshape(2 * T, 512), Wq, kt, vt, Wo)
```

```python
import functools

import jax
import jax.numpy as jnp
from jax import lax
from jax.experimental import pallas as pl
from jax.experimental.pallas import tpu as pltpu

MESH = pl.DeviceIdType.MESH
F32 = jnp.float32
BF16 = jnp.bfloat16
NEG = -1e30
QSCALE = 0.125 * 1.4426950408889634
T = 128
G = 32
A, B, C, D = 0, 1, 2, 3
NN = ((1,), (0,))
NT = ((1,), (1,))

X_ROWS = 48
W_ROWS = 64
HALF = 64
D_SPLIT = 80
HEAD = {(1, 0): 32, (2, 3): 16, (2, 1): 32}

(S_KG, S_VG, S_Q0, S_Q1, S_QG, S_STAT, S_C0, S_C1, S_C2, S_C3, S_C4, S_GS, S_GC0, S_GC1, S_GC2,
 S_HEAD, S_X, S_W, S_K2, S_V2, S_KV) = range(21)
N_RECV = S_KV + 16
N_SEND = 25
N_LOAD = 17


def _sum(xs):
    return functools.reduce(jnp.add, xs)


def _max(xs):
    return functools.reduce(jnp.maximum, xs)


def _iota(shape, dim):
    return lax.broadcasted_iota(jnp.int32, shape, dim)


def _f32(v):
    return v.astype(F32)


def _dot(a, w, dims=NN):
    return lax.dot_general(a, w, (dims, ((), ())), preferred_element_type=F32)


def _dots(lhss, ws, nsplit=None):
    nsplit = nsplit or {1: 4, 2: 2, 3: 4, 4: 1}[len(ws)]
    n = lhss[0].shape[0] // nsplit
    outs = [[] for _ in ws]
    for c in range(nsplit):
        for out, a, (w, dims) in zip(outs, lhss, ws):
            out.append(_dot(a[c * n:(c + 1) * n], w, dims))
    return [o[0] if nsplit == 1 else jnp.concatenate(o, axis=0) for o in outs]


def _pv(ps, vs, nsplit=None):
    return _sum(_dots(ps, vs, nsplit))


def _probs(q2, blocks, nsplit=None):
    ss = _dots([q2] * len(blocks), [k for k, _ in blocks], nsplit)
    ss = [s if mask is None else jnp.where(mask, s, NEG) for s, (_, mask) in zip(ss, blocks)]
    m = jnp.max(_max(ss), axis=1, keepdims=True)
    ps = [jnp.exp2(s - m) for s in ss]
    l = jnp.sum(_sum(ps), axis=1, keepdims=True)
    return [p.astype(BF16) for p in ps], 1.0 / l, m + jnp.log2(l)


def _stack(tile):
    lo = _iota(tile.shape, 1) < 64
    z = jnp.zeros_like(tile)
    return jnp.concatenate([jnp.where(lo, tile, z), jnp.where(lo, z, tile)], axis=0)


def _pair(h0, h1):
    n = h0.shape[0]
    return jnp.where(_iota((n, T), 1) < 64, jnp.broadcast_to(h0, (n, T)), jnp.broadcast_to(h1, (n, T)))


def _unstack(o):
    n = o.shape[0] // 2
    return _pair(o[:n], o[n:])


def _rows2(o, r0, r1):
    n = o.shape[0] // 2
    return jnp.concatenate([o[r0:r1], o[n + r0:n + r1]], axis=0)


def _diag(n, lane0):
    return _iota((n, T), 1) == _iota((n, T), 0) + lane0


def _rows_of_transpose(tile, r0, n):
    return _dot(_diag(n, r0).astype(BF16), tile, NT).astype(BF16)


def _col_to_row(col, lane0):
    n = col.shape[0]
    return jnp.sum(jnp.where(_diag(n, lane0), jnp.broadcast_to(col, (n, T)), 0.0), axis=0, keepdims=True)


def _row_to_col(row, n, lane0):
    return jnp.sum(jnp.where(_diag(n, lane0), jnp.broadcast_to(row, (n, T)), 0.0), axis=1, keepdims=True)


def _merge_weights(lses):
    mx = _max(lses)
    es = [jnp.exp2(e - mx) for e in lses]
    inv = 1.0 / _sum(es)
    return [e * inv for e in es]


def _lane_row(n, row0):
    r = _iota((2 * n, T), 0)
    return _iota((2 * n, T), 1), jnp.where(r < n, r, r - n) + row0


def _global_mask(g):
    lane = _iota((2 * T, T), 1)
    return (lane >= G * g) & (lane < G * g + G)


def _pad_rows(v, before, after):
    parts = [jnp.zeros((before, T), v.dtype)] * bool(before) + [v] + [jnp.zeros((after, T), v.dtype)] * bool(after)
    return jnp.concatenate(parts, axis=0)


def _program(p, bar, x_hbm, wq_hbm, kt_hbm, vt_hbm, wo_hbm, out_ref,
             x32, wq32, wo32, wob, kv32, kv_own, kv_left, kv_right, kv_glob, q_own, q_in, q_glob,
             ctx_in, ctx_out, stat_in, stat_out, glob_ctx, glob_stat, head32, relay, v_keys,
             load_sem, send_sem, recv_sem, ready):
    kv_bufs = {"O": kv_own, "L": kv_left, "R": kv_right}

    def signal(sem, to):
        pl.semaphore_signal(sem, inc=1, device_id=(to,), device_id_type=MESH)

    for to in {0: (1, 3), 1: (2,), 2: (3,), 3: (0, 2)}[p]:
        signal(bar, to)

    loads, started, pending = {}, {"load": 0, "send": 0}, []

    def load(name, src, dst):
        loads[name] = pltpu.make_async_copy(src, dst, load_sem.at[started["load"]])
        started["load"] += 1
        loads[name].start()

    def load_kv(kind, g, r0=0, r1=T):
        load((kind, g, r0), (kt_hbm, vt_hbm)[kind].at[pl.ds(g * T + r0, r1 - r0)],
             kv32.at[kind, g, pl.ds(r0, r1 - r0)])

    def load_x(b):
        load(("x", b), x_hbm.at[pl.ds(b * T, T)], x32.at[pl.ds(b * T, T)])

    def load_wq(hp):
        load(("wq", hp), wq_hbm.at[:, pl.ds(hp * T, T)], wq32.at[hp])

    def wait(*names):
        for name in names:
            loads.pop(name).wait()

    def send(src, dst, slot, to):
        c = pltpu.make_async_remote_copy(src, dst, send_sem.at[started["send"]], recv_sem.at[slot],
                                         device_id=(to,), device_id_type=MESH)
        started["send"] += 1
        c.start()
        pending.append(c)
        return c

    def drain(keep=()):
        for c in pending:
            if not any(c is k for k in keep):
                c.wait_send()
        pending[:] = keep

    def recv(dst, slot):
        pltpu.make_async_remote_copy(dst, dst, send_sem.at[0], recv_sem.at[slot],
                                     device_id=(0,), device_id_type=MESH).wait_recv()

    def rows(r0, r1):
        return pl.ds(r0, r1 - r0)

    def convert(kind, g, r0=0, r1=T):
        wait((kind, g, r0))
        kv_own[kind, g, r0:r1, :] = kv32[kind, g, r0:r1, :].astype(BF16)

    def kv_slot(side, kind, g):
        return S_KV + (0 if side == "L" else 8) + kind * 4 + g

    def send_kv(kind, g, to, r0=0, r1=T, slot=None):
        side = "R" if to < p else "L"
        send(kv_own.at[kind, g, rows(r0, r1)], kv_bufs[side].at[kind, g, rows(r0, r1)],
             kv_slot(side, kind, g) if slot is None else slot, to)

    def send_head(g, to):
        n = HEAD[p, to]
        send(kt_hbm.at[pl.ds(g * T, n)], head32.at[pl.ds(0, n)], S_HEAD, to)

    def recv_kv(side, kind, g, r0=0, r1=T, slot=None):
        recv(kv_bufs[side].at[kind, g, rows(r0, r1)], kv_slot(side, kind, g) if slot is None else slot)

    got = set()

    def recv_k(side, g):
        if (side, 0, g) in got:
            return
        got.add((side, 0, g))
        r = 0
        if (p, side, g) in ((0, "R", A), (3, "L", A), (1, "R", C)):
            r = HEAD[p + (1 if side == "R" else -1), p]
            recv(head32.at[pl.ds(0, r)], S_HEAD)
            kv_bufs[side][0, g, 0:r, :] = head32[0:r, :].astype(BF16)
            if p != 0:
                recv_kv(side, 0, g, r, HALF, S_K2)
                r = HALF
        recv_kv(side, 0, g, r)

    def recv_v(side, g):
        if (side, 1, g) in got:
            return
        got.add((side, 1, g))
        r = T
        if (p, side, g) == (1, "L", A):
            r = T - X_ROWS
            recv_kv(side, 1, g, r, T, S_X)
        recv_kv(side, 1, g, 0, r)

    def send_ctx(i, r0, r1, slot, to):
        return send(ctx_out.at[i, rows(r0, r1)], ctx_in.at[i, rows(r0, r1)], slot, to)

    def recv_ctx(i, r0, r1, slot):
        recv(ctx_in.at[i, rows(r0, r1)], slot)

    relay_x, relay_w = relay.at[pl.ds(0, X_ROWS)], relay.at[pl.ds(0, W_ROWS)]
    glob3 = [kv_glob.at[kind, pl.ds(0, 3 * G)] for kind in range(2)]

    def k_of(side, g):
        return (kv_glob[0], NT) if side == "G" else (kv_bufs[side][0, g], NN)

    def v_of(side, g):
        if side == "G":
            return kv_glob[1], NN
        key_major = (p + {"O": 0, "L": -1, "R": 1}[side], g) == (2, C)
        return kv_bufs[side][1, g], (NN if key_major else NT)

    def q_proj(groups):
        for g in groups:
            b, hp = divmod(g, 2)
            q = _dot(x32[b * T:(b + 1) * T, :].astype(BF16), wq32[hp].astype(BF16))
            q_own[g] = (q * QSCALE).astype(BF16)

    def pack_global(kind):
        for g in range(4):
            kv_glob[kind, G * g:G * g + G, :] = _rows_of_transpose(kv_own[kind, g], 0, G)

    def wo_prep():
        wait("wo")
        wob[...] = wo32[...].astype(BF16)

    def proj(g, ctx):
        hp = g % 2
        return _dot(ctx.astype(BF16), wob[hp * T:(hp + 1) * T, :])

    def scores(g, sides, early):
        for s in sides:
            if s in "LR":
                recv_k(s, g)
        for s in early:
            if s in "LR":
                recv_v(s, g)
        lane, row = _lane_row(T, 0)
        mask = {"O": None, "G": _global_mask(g),
                "L": (lane >= row) | (lane < G) if p == 1 else lane >= row,
                "R": (lane <= row) | (row < G) if p == 0 else lane <= row}
        ps, linv, lse = _probs(_stack(q_own[g]), [(k_of(s, g), mask[s]) for s in sides])
        ps = dict(zip(sides, ps))
        o = _pv([ps.pop(s) for s in early], [v_of(s, g) for s in early])
        return g, ps, o, linv, lse

    def values(st):
        g, ps, o, linv, _ = st
        for s in ps:
            if s == "G":
                recv(glob3[1], S_VG)
            else:
                recv_v(s, g)
        if ps:
            o = o + _pv(list(ps.values()), [v_of(s, g) for s in ps])
        return _unstack(o * linv)

    written = set()

    def finish(st, r0=0):
        g, ctx = st[0], values(st)
        if g // 2 in written:
            out_ref[g // 2, r0:, :] += proj(g, ctx[r0:])
        else:
            out_ref[g // 2, r0:, :] = proj(g, ctx[r0:])
            written.add(g // 2)
        return ctx

    def part_scores(q_tile, blocks, nsplit=None):
        return _probs(_stack(q_tile), [(k_of(s, g), mask) for s, g, mask in blocks], nsplit)

    def part_values(st, blocks, nsplit=None):
        return _unstack(_pv(st[0], [v_of(s, g) for s, g, _ in blocks], nsplit) * st[1]).astype(BF16)

    def serve(blocks, to):
        recv(q_in.at[0], S_Q0)
        st = part_scores(q_in[0], blocks)
        ctx_out[0] = part_values(st, blocks)
        for h in range(2):
            stat_out[h:h + 1, :] = _col_to_row(st[2][T * h:T * h + T], 0)
        return [send(stat_out.at[pl.ds(0, 2)], stat_in.at[pl.ds(0, 2)], S_STAT, to),
                send_ctx(0, 0, HALF, S_C0, to), send_ctx(0, HALF, T, S_C1, to)]

    def remote_lse(i=0):
        return _pair(_row_to_col(stat_in[2 * i:2 * i + 1, :], T, 0),
                     _row_to_col(stat_in[2 * i + 1:2 * i + 2, :], T, 0))

    if p == 0:
        load_x(1); load_wq(0)
        for g in (C, D, A, B):
            load_kv(0, g)
        load_wq(1)
        for g in (C, D, A, B):
            load_kv(1, g)
        load_x(0)
        load("wo", wo_hbm, wo32)
        wait(("x", 1), ("wq", 0))
        q_proj([C])
        for g in (C, D, A, B):
            convert(0, g)
        pack_global(0)
        pl.semaphore_wait(ready, 1)
        send(q_own.at[C], q_in.at[0], S_Q0, 1)
        pl.semaphore_wait(bar, 1)
        send(kv_glob.at[0], kv_glob.at[0], S_KG, 3)
        wait(("wq", 1))
        q_proj([D])
        send(q_own.at[D], q_in.at[1], S_Q1, 1)
        send_kv(0, C, 1)
        for g in (C, D, A, B):
            convert(1, g)
        send_kv(1, C, 1); send_kv(0, D, 1); send_kv(1, D, 1)
        send_kv(0, A, 1); send_kv(1, A, 1, 0, T - X_ROWS)
        pack_global(1)
        send(kv_glob.at[1], kv_glob.at[1], S_VG, 3)
        wait(("x", 0))
        q_proj([A, B])
        for g in range(4):
            q_glob[g] = q_own[g, 0:G, :]
        send(q_glob, q_glob, S_QG, 3)
        send(kv_own.at[1, A, rows(T - X_ROWS, T)], relay_x, S_X, 3)
        loc, lse = {}, {}
        for g in (C, D):
            st = scores(g, "O", "O")
            loc[g], lse[g] = values(st), _unstack(st[4])
        wo_prep()
        for g in (A, B):
            st = scores(g, "OR", "O")
            loc[g], lse[g] = finish(st, G)[0:G], _unstack(_rows2(st[4], 0, G))
        lane, row = _lane_row(T, 0)
        keep = serve([("O", B, (lane >= row) | (lane < G))], 1)
        recv(relay_w, S_W)
        send(relay_w, kv_left.at[1, C, rows(T - W_ROWS, T)], S_W, 3)
        recv(glob_stat, S_GS); recv(stat_in, S_STAT)
        w3, w1 = {}, {}
        for g in range(4):
            e3 = _unstack(_row_to_col(glob_stat[g // 2:g // 2 + 1, :], 2 * G, 64 * (g % 2)))
            if g < C:
                wl, w3[g] = _merge_weights([lse[g], e3])
            else:
                e1 = remote_lse(g - C)
                wa, wb = _merge_weights([lse[g][G:], e1[G:]])
                wga, wgb, w3[g] = _merge_weights([lse[g][0:G], e1[0:G], e3])
                wl = jnp.concatenate([wga, wa], axis=0)
                w1[g] = jnp.concatenate([wgb, wb], axis=0)
            loc[g] = loc[g] * wl
        drain(keep)

        def merged(g, r0, r1):
            return loc[g][r0:r1] + w1[g][r0:r1] * _f32(ctx_in[g - C, r0:r1, :])

        def from3(g):
            return w3[g] * _f32(glob_ctx[g])

        recv_ctx(0, G, T, S_C0); recv_ctx(0, 0, G, S_C2)
        recv(glob_ctx.at[A], S_GC0); recv(glob_ctx.at[pl.ds(C, 2)], S_GC1); recv_ctx(1, G, D_SPLIT, S_C1)
        o_even = proj(A, jnp.concatenate([loc[A] + from3(A), merged(C, 0, G) + from3(C), merged(C, G, T)], axis=0))
        out_ref[1, G:D_SPLIT, :] = o_even[2 * G:G + D_SPLIT] + proj(D, merged(D, G, D_SPLIT))
        o_glob, o_c = o_even[0:2 * G], o_even[G + D_SPLIT:]
        recv(glob_ctx.at[B], S_GC2); recv_ctx(1, 0, G, S_C3)
        o_glob = o_glob + proj(B, jnp.concatenate([loc[B] + from3(B), merged(D, 0, G) + from3(D)], axis=0))
        out_ref[0, 0:G, :] = o_glob[0:G]
        out_ref[1, 0:G, :] = o_glob[G:]
        recv_ctx(1, D_SPLIT, T, S_C4)
        out_ref[1, D_SPLIT:, :] = o_c + proj(D, merged(D, D_SPLIT, T))

    elif p == 1:
        h10 = HEAD[1, 0]
        pl.semaphore_wait(bar, 1)
        signal(ready, 0)
        send_head(A, 0)
        load_kv(0, A, h10)
        load_kv(1, A)
        for g in (B, D):
            load_kv(0, g); load_kv(1, g)
        load_kv(0, A, 0, h10)
        load_kv(0, C); load_kv(1, C)
        load_x(0); load_wq(1); load_x(1); load_wq(0)
        load("wo", wo_hbm, wo32)
        convert(0, A, h10); send_kv(0, A, 0, h10)
        for kind, g in ((1, A), (0, B), (1, B)):
            convert(kind, g)
            send_kv(kind, g, 0)
        convert(0, D); convert(1, D)
        convert(0, A, 0, h10); convert(0, C); convert(1, C)
        pl.semaphore_wait(ready, 1)
        for g in (D, A, B, C):
            send_kv(0, g, 2); send_kv(1, g, 2)
        wait(("x", 0), ("wq", 1))
        q_proj([B])
        send(q_own.at[B], q_in.at[0], S_Q0, 0)
        wait(("x", 1), ("wq", 0))
        q_proj([C, D, A])
        recv(q_in.at[0], S_Q0); recv_k("R", C); recv(q_in.at[1], S_Q1)
        lane, row = _lane_row(T - G, G)
        hi, lo = {}, {}
        for g in (C, D):
            blocks = [("O", g, lane <= row)]
            hi[g] = part_scores(q_in[g - C, G:, :], blocks, 2)
            ctx_out[g - C, G:, :] = part_values(hi[g], blocks, 2)
        lo_blocks = {g: [("O", g, None), ("R", g, None)] for g in (C, D)}
        lo[C] = part_scores(q_in[0, 0:G, :], lo_blocks[C], 2)
        recv_v("R", C)
        send(kv_right.at[1, C, rows(T - W_ROWS, T)], relay_w, S_W, 0)
        send_ctx(0, G, T, S_C0, 0)
        wo_prep()
        st_c = scores(C, "OLR", "OR")
        recv_k("R", D)
        lo[D] = part_scores(q_in[1, 0:G, :], lo_blocks[D], 2)
        ctx_out[0, 0:G, :] = part_values(lo[C], lo_blocks[C], 2)
        o = _pv([lo[D][0][0]], [v_of("O", D)])
        for g in (C, D):
            for h in range(2):
                i = 2 * (g - C) + h
                stat_out[i:i + 1, :] = (_col_to_row(lo[g][2][G * h:G * h + G], 0)
                                        + _col_to_row(hi[g][2][(T - G) * h:(T - G) * (h + 1)], G))
        send(stat_out, stat_in, S_STAT, 0)
        send_ctx(0, 0, G, S_C2, 0); send_ctx(1, G, D_SPLIT, S_C1, 0)
        recv_v("R", D)
        o = o + _pv([lo[D][0][1]], [v_of("R", D)])
        ctx_out[1, 0:G, :] = _unstack(o * lo[D][1]).astype(BF16)
        send_ctx(1, 0, G, S_C3, 0); send_ctx(1, D_SPLIT, T, S_C4, 0)
        finish(st_c)
        finish(scores(D, "OLR", "OR"))
        _, ps, o, linv, lse_b = scores(B, "OR", "O")
        st_a = scores(A, "OLR", "O")
        recv(stat_in.at[pl.ds(0, 2)], S_STAT)
        recv_v("L", A); recv_v("R", A)
        wa, wb = _merge_weights([_unstack(lse_b), remote_lse()])
        finish(st_a)
        drain()
        recv_ctx(0, 0, HALF, S_C0); recv_kv("R", 1, B, 0, HALF, S_V2)
        o = o + _pv([ps["R"]], [(_pad_rows(kv_right[1, B, 0:HALF, :], 0, T - HALF), NN)])
        out_ref[0, 0:HALF, :] += proj(B, _unstack(_rows2(o * linv, 0, HALF)) * wa[:HALF]
                                      + wb[:HALF] * _f32(ctx_in[0, 0:HALF, :]))
        o, linv, p_hi = _rows2(o, HALF, T), _rows2(linv, HALF, T), _rows2(ps["R"], HALF, T)
        recv_ctx(0, HALF, T, S_C1); recv_kv("R", 1, B, HALF, T)
        o = o + _pv([p_hi], [(_pad_rows(kv_right[1, B, HALF:, :], HALF, 0), NN)])
        out_ref[0, HALF:, :] += proj(B, _unstack(o * linv) * wa[HALF:] + wb[HALF:] * _f32(ctx_in[0, HALF:, :]))

    elif p == 2:
        h23, h21 = HEAD[2, 3], HEAD[2, 1]
        load_kv(0, A, h23, HALF)
        pl.semaphore_wait(bar, 2)
        send_head(A, 3)
        send_head(C, 1)
        signal(ready, 1)
        load_kv(0, C, h21, HALF); load_kv(0, A, HALF); load_kv(0, C, HALF)
        load_kv(1, A); load_kv(1, C)
        for kind in range(2):
            load_kv(kind, B); load_kv(kind, D)
        load_kv(0, A, 0, h23); load_kv(0, C, 0, h21)
        load_x(1); load_wq(1); load_wq(0); load_x(0)
        load("wo", wo_hbm, wo32)
        kv_glob[:, 3 * G:, :] = jnp.zeros((2, G, T), BF16)
        convert(0, A, h23, HALF); send_kv(0, A, 3, h23, HALF, S_K2)
        convert(0, C, h21, HALF); send_kv(0, C, 1, h21, HALF, S_K2)
        convert(0, A, HALF); send_kv(0, A, 3, HALF)
        convert(0, C, HALF); send_kv(0, C, 1, HALF)
        convert(1, A); send_kv(1, A, 3)
        wait((1, C, 0))
        v_c = kv32[1, C].astype(BF16)
        for r in range(0, T, 32):
            kv_own[1, C, r:r + 32, :] = _rows_of_transpose(v_c, r, 32)
        send_kv(1, C, 1)
        for kind in range(2):
            convert(kind, B); send_kv(kind, B, 3)
            convert(kind, D); send_kv(kind, D, 1)
        convert(0, A, 0, h23); convert(0, C, 0, h21)
        send_kv(0, A, 1); send_kv(0, B, 1); send_kv(1, A, 1)
        wait(("x", 1), ("wq", 1))
        q_proj([D])
        send(q_own.at[D], q_in.at[0], S_Q0, 3)
        send_kv(0, D, 3); send_kv(0, C, 3); send_kv(1, D, 3); send_kv(1, C, 3, 0, T - W_ROWS)
        wait(("wq", 0), ("x", 0))
        q_proj([C, A, B])
        st = scores(D, "OL", "O")
        ctx_d, lse_d = values(st), _unstack(st[4])
        wo_prep()
        for r in range(0, T, 32):
            v_keys[r:r + 32, :] = _rows_of_transpose(kv_own[1, B], r, 32)
        recv(glob3[0], S_KG)
        finish(scores(A, "OGLR", "OR"))
        recv_k("R", B)
        recv(relay_x, S_X)
        send(relay_x, kv_left.at[1, A, rows(T - X_ROWS, T)], S_X, 1)
        send(v_keys.at[rows(0, HALF)], kv_right.at[1, B, rows(0, HALF)], S_V2, 1)
        send(v_keys.at[rows(HALF, T)], kv_right.at[1, B, rows(HALF, T)], kv_slot("R", 1, B), 1)
        finish(scores(B, "OGLR", "OG"))
        st = scores(C, "OGLR", "OG")
        drain()
        recv(stat_in.at[pl.ds(0, 2)], S_STAT)
        recv_v("L", C); recv_v("R", C)
        wa, wb = _merge_weights([lse_d, remote_lse()])
        ctx_d = ctx_d * wa
        finish(st)
        for r0, r1, slot in ((0, HALF, S_C0), (HALF, T, S_C1)):
            recv_ctx(0, r0, r1, slot)
            out_ref[1, r0:r1, :] += proj(D, ctx_d[r0:r1] + wb[r0:r1] * _f32(ctx_in[0, r0:r1, :]))

    else:
        for g in (A, B, C, D):
            load_kv(0, g); load_kv(1, g)
        load_x(0); load_wq(0); load_wq(1); load_x(1)
        load("wo", wo_hbm, wo32)
        for g in (A, B, C, D):
            convert(0, g); convert(1, g)
        pl.semaphore_wait(bar, 2)
        send_kv(0, A, 2); send_kv(1, A, 2)
        recv(kv_glob.at[0], S_KG)
        send(glob3[0], glob3[0], S_KG, 2)
        wait(("x", 0), ("wq", 0), ("wq", 1), ("x", 1))
        q_proj([A, B, C, D])
        recv(kv_glob.at[1], S_VG)
        send(glob3[1], glob3[1], S_VG, 2)
        send_kv(0, B, 2)
        wo_prep()
        finish(scores(A, "OGL", "OGL"))
        recv(relay_x, S_X)
        send(relay_x, relay_x, S_X, 2)
        send_kv(1, B, 2); send_kv(0, C, 2); send_kv(1, C, 2)
        recv(q_glob, S_QG)
        recv_k("L", B)
        blocks = {g: [("O", g, None)] + [("L", g, None)] * (g < C) for g in range(4)}
        sts = {g: part_scores(q_glob[g], blocks[g], 1 if g < C else 2) for g in range(4)}
        for b in range(2):
            glob_stat[b:b + 1, :] = _col_to_row(sts[2 * b][2], 0) + _col_to_row(sts[2 * b + 1][2], 64)
        for g in (A, C, D):
            glob_ctx[g] = part_values(sts[g], blocks[g], 1)
        send(glob_stat, glob_stat, S_GS, 0)
        send(glob_ctx.at[A], glob_ctx.at[A], S_GC0, 0)
        send(glob_ctx.at[pl.ds(C, 2)], glob_ctx.at[pl.ds(C, 2)], S_GC1, 0)
        st = scores(B, "OGL", "OG")
        recv_v("L", B)
        glob_ctx[B] = part_values(sts[B], blocks[B], 2)
        send(glob_ctx.at[B], glob_ctx.at[B], S_GC2, 0)
        finish(st)
        lane, row = _lane_row(T, 0)
        keep = serve([("O", D, lane <= row), ("G", D, _global_mask(D))], 2)
        st_d = scores(D, "OGL", "OG")
        n = T - W_ROWS
        recv_kv("L", 1, C, n, T, S_W)
        _, ps, o, linv, _ = scores(C, "OGL", "OG")
        o = o + _pv([ps["L"]], [(_pad_rows(kv_left[1, C, n:, :], n, 0), NN)])
        o_hi = proj(C, _unstack(_rows2(o * linv, n, T)))
        o, linv, p_lo = _rows2(o, 0, n), _rows2(linv, 0, n), _rows2(ps["L"], 0, n)
        drain(keep)
        o_d = proj(D, values(st_d))
        out_ref[1, n:, :] = o_d[n:] + o_hi
        o_d = o_d[:n]
        drain()
        recv_kv("L", 1, C, 0, n)
        o = o + _pv([p_lo], [(_pad_rows(kv_left[1, C, 0:n, :], 0, W_ROWS), NN)])
        out_ref[1, 0:n, :] = o_d + proj(C, _unstack(o * linv))

    drain()
    assert not loads and started["load"] <= N_LOAD and started["send"] <= N_SEND


def pallas_dist_sparse_attn_localglobal_qseq_kvseq_b2_sq128_skv128_hq4_dh64_kernel(
    x: jax.Array,
    Wq: jax.Array,
    K_ext: jax.Array,
    V_ext: jax.Array,
    Wo: jax.Array,
):
    kt = jnp.transpose(K_ext, (0, 2, 3, 1)).reshape(4 * T, T)
    vt = jnp.transpose(V_ext, (0, 2, 3, 1)).reshape(4 * T, T)

    def body(*refs):
        my = lax.axis_index("i")
        bar = pltpu.get_barrier_semaphore()
        for p in range(4):
            pl.when(my == p)(functools.partial(_program, p, bar, *refs))

    vmem = pltpu.VMEM
    return pl.pallas_call(
        body,
        out_shape=jax.ShapeDtypeStruct((2, T, 512), F32),
        in_specs=[pl.BlockSpec(memory_space=pl.ANY)] * 5,
        out_specs=pl.BlockSpec(memory_space=pltpu.VMEM),
        scratch_shapes=[
            vmem((2 * T, 512), F32),
            vmem((2, 512, T), F32),
            vmem((2 * T, 512), F32),
            vmem((2 * T, 512), BF16),
            vmem((2, 4, T, T), F32),
            vmem((2, 4, T, T), BF16),
            vmem((2, 4, T, T), BF16),
            vmem((2, 4, T, T), BF16),
            vmem((2, T, T), BF16),
            vmem((4, T, T), BF16),
            vmem((2, T, T), BF16),
            vmem((4, G, T), BF16),
            vmem((2, T, T), BF16),
            vmem((2, T, T), BF16),
            vmem((4, T), F32),
            vmem((4, T), F32),
            vmem((4, G, T), BF16),
            vmem((2, T), F32),
            vmem((32, T), F32),
            vmem((64, T), BF16),
            vmem((T, T), BF16),
            pltpu.SemaphoreType.DMA((N_LOAD,)),
            pltpu.SemaphoreType.DMA((N_SEND,)),
            pltpu.SemaphoreType.DMA((N_RECV,)),
            pltpu.SemaphoreType.REGULAR,
        ],
        compiler_params=pltpu.CompilerParams(collective_id=0, disable_semaphore_checks=True),
    )(x.reshape(2 * T, 512), Wq, kt, vt, Wo)
```
